```python
import numpy as np

kernel_name = "dist_ar_i_i_m2048_n512"

def setup_inputs():
    return {"x": np.random.randn(8192, 512).astype(np.float32)}

def reference(x: np.ndarray) -> np.ndarray:
    return x.reshape(4, 2048, 512).sum(axis=0)
```

```python
import jax
import jax.numpy as jnp
from jax import lax
from jax.experimental import pallas as pl
from jax.experimental.pallas import tpu as pltpu

M, N = 2048, 512
Q = M // 4
CH1 = (16, 16, 32, 64, 128, 128, 128)
CH2 = (128, 128, 128, 128)
CH3 = (128, 128, 128, 64, 32, 16, 16)


def _offs(ch):
    out, o = [], 0
    for c in ch:
        out.append((o, c)); o += c
    assert o == Q
    return out


def pallas_dist_ar_i_i_m2048_n512_kernel(x):
    c1, c2, c3 = _offs(CH1), _offs(CH2), _offs(CH3)
    n1, n2, n3 = len(c1), len(c2), len(c3)

    def body(x_hbm, o_hbm, xs, xk, s1, r1, s2, r2, s3, r3, ok, og,
             ld_s, ld_k, snd1, rcv1, snd2, rcv2, snd3, rcv3, st_k, st_g):
        p = lax.axis_index("i")
        nbr = (p ^ 1, p ^ 3)
        bit = ((p ^ (p >> 1)) & 1, p >> 1)
        keep = [pl.multiple_of(h * 2 * Q + bit[h] * Q, Q) for h in range(2)]
        give = [pl.multiple_of(h * 2 * Q + (1 - bit[h]) * Q, Q) for h in range(2)]

        bar = pltpu.get_barrier_semaphore()
        for h in range(2):
            pl.semaphore_signal(bar, 1, device_id=(nbr[h],), device_id_type=pl.DeviceIdType.MESH)

        def rdma(src, dst, ss, rs, h):
            return pltpu.make_async_remote_copy(src, dst, ss, rs, device_id=(nbr[h],),
                                                device_id_type=pl.DeviceIdType.MESH)

        lds = {}
        for i, (o, c) in enumerate(c1):
            for h in range(2):
                lds[h, i] = pltpu.make_async_copy(x_hbm.at[pl.ds(give[h] + o, c)], xs.at[h, pl.ds(o, c)], ld_s.at[h * n1 + i])
                lds[h, i].start()
        ldk = [pltpu.make_async_copy(x_hbm.at[pl.ds(keep[h], Q)], xk.at[h], ld_k.at[h]) for h in range(2)]
        for d in ldk:
            d.start()

        d1, d2, d3, sts = {}, {}, {}, []
        for i, (o, c) in enumerate(c1):
            sl = pl.ds(o, c)
            for h in range(2):
                lds[h, i].wait()
                s1[h, sl] = xs[h, sl].astype(jnp.bfloat16)
            if i == 0:
                pl.semaphore_wait(bar, 2)
            for h in range(2):
                d1[h, i] = rdma(s1.at[h, sl], r1.at[h, sl], snd1.at[h * n1 + i], rcv1.at[h * n1 + i], h)
                d1[h, i].start()
        for d in ldk:
            d.wait()
        k = 0
        for i, (o, c) in enumerate(c2):
            sl = pl.ds(o, c)
            while k < n1 and c1[k][0] < o + c:
                for h in range(2):
                    d1[h, k].wait_recv()
                k += 1
            for h in range(2):
                t = xk[h, sl] + r1[h, sl].astype(jnp.float32)
                s2[h, sl] = t.astype(jnp.bfloat16)
                d2[h, i] = rdma(s2.at[h, sl], r2.at[h, sl], snd2.at[h * n2 + i], rcv2.at[h * n2 + i], 1 - h)
                d2[h, i].start()
        k = 0
        for i, (o, c) in enumerate(c3):
            sl = pl.ds(o, c)
            while k < n2 and c2[k][0] < o + c:
                for h in range(2):
                    d2[h, k].wait_recv()
                k += 1
            for h in range(2):
                t = (s2[h, sl].astype(jnp.float32) + r2[h, sl].astype(jnp.float32)).astype(jnp.bfloat16)
                s3[h, sl] = t
                d3[h, i] = rdma(s3.at[h, sl], r3.at[h, sl], snd3.at[h * n3 + i], rcv3.at[h * n3 + i], h)
                d3[h, i].start()
                ok[h, sl] = t.astype(jnp.float32)
                st = pltpu.make_async_copy(ok.at[h, sl], o_hbm.at[pl.ds(keep[h] + o, c)], st_k.at[h * n3 + i])
                st.start(); sts.append(st)
        for i, (o, c) in enumerate(c3):
            sl = pl.ds(o, c)
            for h in range(2):
                d3[h, i].wait_recv()
                og[h, sl] = r3[h, sl].astype(jnp.float32)
                st = pltpu.make_async_copy(og.at[h, sl], o_hbm.at[pl.ds(give[h] + o, c)], st_g.at[h * n3 + i])
                st.start(); sts.append(st)
        for d in (*d1.values(), *d2.values(), *d3.values()):
            d.wait_send()
        for st in sts:
            st.wait()

    f32 = lambda: pltpu.VMEM((2, Q, N), jnp.float32)
    b16 = lambda: pltpu.VMEM((2, Q, N), jnp.bfloat16)
    sem = lambda n: pltpu.SemaphoreType.DMA((2 * n,))
    return pl.pallas_call(
        body,
        out_shape=pltpu.HBM((M, N), jnp.float32),
        in_specs=[pl.BlockSpec(memory_space=pltpu.HBM)],
        out_specs=pl.BlockSpec(memory_space=pltpu.HBM),
        scratch_shapes=[f32(), f32(), b16(), b16(), b16(), b16(), b16(), b16(), f32(), f32(),
                        sem(n1), sem(1), sem(n1), sem(n1), sem(n2), sem(n2), sem(n3), sem(n3), sem(n3), sem(n3)],
        compiler_params=pltpu.CompilerParams(collective_id=0, vmem_limit_bytes=64 * 2**20),
    )(x)
```

```python
import contextlib
import jax
import jax.numpy as jnp
from jax import lax
from jax.experimental import pallas as pl
from jax.experimental.pallas import tpu as pltpu

M, N = 2048, 512
H = M // 2
EXTRA = 0
PH1 = (16, 48, ((64,),), ((64, 64),), ((64,) * 4,))
PH2 = (((64,) * 4,), ((64,) * 4,))
PH3 = (((64,) * 4,), ((64, 64), (64,), (64,)))
LATE = 2
KEEP_AT = 3
SOLO = ()
XAT = (99, 99, 1)
UNROLL = True
CP = dict(disable_semaphore_checks=True)
SCOPES = False

I32 = jnp.int32
srl, sll = lax.shift_right_logical, lax.shift_left


def _scope(n):
    return jax.named_scope('z' + n) if SCOPES else contextlib.nullcontext()


def _i(v):
    return I32(v - (1 << 32) if v >= (1 << 31) else v)


def _splat(v):
    return jnp.full((8, 128), _i(v), I32)


def _to_words(v):
    w = pltpu.bitcast(v.astype(jnp.bfloat16), I32)
    return [w[8 * i:8 * i + 8, 128 * j:128 * j + 128] for i in range(w.shape[0] // 8) for j in range(4)]


def _from_words(ws):
    rows = [jnp.concatenate(ws[i:i + 4], axis=1) for i in range(0, len(ws), 4)]
    return pltpu.bitcast(jnp.concatenate(rows, axis=0), jnp.bfloat16)


def _bitrev(v):
    for s, m in ((1, 0x55555555), (2, 0x33333333), (4, 0x0F0F0F0F), (8, 0x00FF00FF)):
        v = (srl(v, I32(s)) & _i(m)) | sll(v & _i(m), I32(s))
    return srl(v, I32(16)) | sll(v, I32(16))


def _first():
    return (lax.broadcasted_iota(I32, (8, 128), 0) == 0) & (lax.broadcasted_iota(I32, (8, 128), 1) == 0)


def _packed(n):
    return -(-11 * n // 16)


def _max_exp(ws):
    es = [w & _i(0x7F807F80) for w in ws]
    es = [jnp.maximum(e, sll(e, I32(16))) for e in es]
    return jnp.maximum(jnp.maximum(es[0], es[1]), jnp.maximum(es[2], es[3]))


def _shr64(hi, lo, n):
    return srl(hi, n), srl(lo, n) | sll(sll(hi, I32(1)), 31 - n)


def _shl64(hi, lo, n):
    return sll(hi, n) | srl(srl(lo, I32(1)), 31 - n), ~sll(~lo, n)


def _encode_group(ws, base, state):
    hi, lo, total, worst = state
    bh, bl = sll(base, I32(23)), sll(base, I32(7))
    ch, cl = bh + _i(1 << 23), bl + _i(1 << 7)
    b2, c2 = bh | bl, ch | cl
    top = _splat(1 << 31)
    acc_h = acc_l = top
    run = _splat(0)
    out = []
    for w in ws:
        eh, el = w & _i(0x7F800000), w & _i(0x00007F80)
        code = (jnp.maximum(eh, bh) | jnp.maximum(el, bl)) - b2
        run = run + srl(c2 - (jnp.minimum(eh, ch) | jnp.minimum(el, cl)), I32(7))
        pos_h, pos_l = srl(run, I32(16)), run & _i(0xFFFF)
        acc_h = acc_h | srl(top, pos_h)
        acc_l = acc_l | srl(top, pos_l)
        out.append((w & _i(0x807F807F)) | code)
    k, m = _packed(len(ws)), _i(0x7C007C00)
    for j, d in enumerate(out[k:]):
        out[2 * j] = out[2 * j] | (sll(d, I32(10)) & m)
        out[2 * j + 1] = out[2 * j + 1] | (sll(d, I32(5)) & m)
        out[k - 1] = out[k - 1] | srl(d & _i(0x80008000), I32(1 + j))
    for acc, pos in ((acc_l, pos_l), (acc_h, pos_h)):
        total = total + pos
        worst = jnp.maximum(worst, pos)
        hi, lo = _shr64(hi, lo, jnp.minimum(pos, 31))
        hi = hi | acc
    return out[:k], (hi, lo, total, worst)


def _encode_finish(gmax, emax, state):
    hi, lo, total, worst = state
    first = _first()
    lead = gmax - emax + jnp.where(first, 9, 0)
    total = total + lead + 1
    worst = jnp.maximum(worst, lead)
    hi, lo = _shr64(hi, lo, jnp.minimum(lead, 31))
    side = hi | jnp.where(first, sll(gmax, I32(23)), 0) | _bitrev(pltpu.roll(lo, 4, 0))
    excess = jnp.maximum(worst - 31, total + pltpu.roll(total, 4, 0) - 64)
    return side, jnp.max(excess.astype(jnp.float32)) > 0


def _decode_start(side, head):
    hi, lo = _shl64(side, _bitrev(pltpu.roll(side, 4, 0)), jnp.where(_first(), 9, 0))
    lead = lax.clz(hi)
    base = srl(head, I32(23)) - 7 - lead
    hi, lo = _shl64(*_shl64(hi, lo, lead), _splat(1))
    return sll(base, I32(23)) | sll(base, I32(7)), (hi, lo)


def _decode_group(ps, n, b2, state):
    hi, lo = state
    k, m = len(ps), _i(0x7C007C00)
    ws = list(ps)
    for j in range(n - k):
        ws.append(srl(ps[2 * j] & m, I32(10)) | srl(ps[2 * j + 1] & m, I32(5))
                  | (sll(ps[k - 1], I32(1 + j)) & _i(0x80008000)))
    es = [b2 + (w & _i(0x03800380)) for w in ws]
    for sh in (23, 7):
        acc, used = hi, lax.population_count(hi)
        for i, w in enumerate(ws):
            esc = (w & _i(7 << sh)) == 0
            z = lax.clz(acc)
            zz = jnp.where(esc, z, 0)
            es[i] = es[i] - sll(zz, I32(sh))
            used = used + zz
            acc = jnp.where(esc, sll(sll(acc, I32(1)), z), acc)
        used = used - lax.population_count(acc)
        hi, lo = acc | srl(srl(lo, I32(1)), 31 - used), ~sll(~lo, used)
    return [(w & _i(0x807F807F)) | e for w, e in zip(ws, es)], (hi, lo)


class _Piece:
    def __init__(self, phase, row, spec, slot, sem):
        self.phase, self.row, self.slot, self.sem = phase, row, slot, sem
        self.coded = not isinstance(spec, int)
        if self.coded:
            self.groups, self.cuts, r, at = [], [], row, slot + 1
            for cut in spec:
                start = slot if not self.cuts else at
                for g in cut:
                    self.groups.append((r, g, at))
                    r, at = r + g, at + _packed(g // 4)
                self.cuts.append((start, at - start, len(self.groups)))
            self.rows = r - row
            self.end = slot + 1 + self.rows // 4
            self.spill = (at, self.end - at)
        else:
            self.rows = spec
            self.end = slot + spec // 4
            self.cuts = [(slot, spec // 4, 0)]
        self.nsem = len(self.cuts) + self.coded


def pallas_dist_ar_i_i_m2048_n512_kernel(x):
    C = (H - EXTRA) // 2
    phs, extra, nslot, nsem = [], [], 0, 0
    for s, specs in enumerate((PH1, PH2, PH3)):
        row, ps = 0, []
        for spec in specs + (((EXTRA,),),) * (EXTRA > 0):
            ps.append(_Piece(s, row, spec, nslot, nsem))
            row, nslot, nsem = row + ps[-1].rows, ps[-1].end, nsem + ps[-1].nsem
        assert row == C + EXTRA
        extra.append(ps.pop() if EXTRA else None)
        phs.append(ps)
    n1, R = len(phs[0]), C + EXTRA

    def body(x_hbm, o_ref, xs, xk, part, wbuf, mbuf, sbuf, rbuf, spilled, ld, snd, rcv, ready):
        p = lax.axis_index("i")
        odd = p & 1
        swap = (p == 3).astype(I32)
        half = (swap, 1 - swap)
        nbr = [p ^ (1 + 2 * half[h]) for h in range(2)]
        bit = [jnp.where(half[h] == 0, (p ^ (p >> 1)) & 1, p >> 1) for h in range(2)]
        keep = [half[h] * H + bit[h] * C for h in range(2)]
        give = [half[h] * H + (1 - bit[h]) * C for h in range(2)]
        xrow = [half[h] * H + 2 * C for h in range(2)]
        mesh = pl.DeviceIdType.MESH

        def rows(base, h, r, n):
            return pl.ds(pl.multiple_of(xrow[h] + (r - C) if r >= C else base[h] + r, 16), n)

        lds = {}
        for i, pc in enumerate(phs[0]):
            for h in range(2):
                lds[h, i] = pltpu.make_async_copy(x_hbm.at[rows(give, h, pc.row, pc.rows)],
                                                  xs.at[h, pl.ds(pc.row, pc.rows)], ld.at[2 * i + h])
        ldk = [pltpu.make_async_copy(x_hbm.at[rows(keep, h, 0, C)], xk.at[h, pl.ds(0, C)], ld.at[2 * n1 + h]) for h in range(2)]
        if EXTRA:
            ldk += [pltpu.make_async_copy(x_hbm.at[rows(keep, h, C, EXTRA)], xk.at[h, pl.ds(C, EXTRA)], ld.at[2 * n1 + 2 + h]) for h in range(2)]

        lds[0, 0].start()
        bar = pltpu.get_barrier_semaphore()

        @pl.when(p != 2)
        def _():
            for h in range(2):
                pl.semaphore_signal(bar, 1, device_id=(nbr[h],), device_id_type=mesh)
        for d in list(lds.values())[1:]:
            d.start()
        with _scope("bar"):
            pl.semaphore_wait(bar, 2 - odd)

        @pl.when(p == 2)
        def _():
            for h in range(2):
                pl.semaphore_signal(ready, 1, device_id=(nbr[h],), device_id_type=mesh)

        def copy(pc, h, k):
            at, n = pc.cuts[k][:2] if k < len(pc.cuts) else pc.spill
            if pc.phase == 2 and not pc.coded:
                src = dst = o_ref.at[rows(keep, h, pc.row, pc.rows)]
            else:
                src, dst = sbuf.at[h, pl.ds(at, n)], rbuf.at[half[h], pl.ds(at, n)]
            j = 2 * (pc.sem + k)
            return pltpu.make_async_remote_copy(src, dst, snd.at[j + h], rcv.at[j + half[h]],
                                                device_id=(nbr[h ^ (pc.phase == 1)],), device_id_type=mesh)

        def get(ref, h, at, n):
            return [ref[h, at + j] for j in range(n)]

        def put(ref, h, at, ws):
            for j, w in enumerate(ws):
                ref[h, at + j] = w

        def stage(h, r, v):
            ws = _to_words(v)
            put(wbuf, h, r // 4, ws)
            put(mbuf, h, r // 16, [_max_exp(ws[j:j + 4]) for j in range(0, len(ws), 4)])

        def over_groups(groups, f, carry):
            i = 0
            while i < len(groups):
                j = i + 1
                while not UNROLL and j < len(groups) and groups[j][1] == groups[i][1]:
                    j += 1
                r, g, at = groups[i]
                if j == i + 1:
                    carry = f(r, g, at, carry)
                else:
                    dr, da = groups[i + 1][0] - r, groups[i + 1][2] - at
                    carry = lax.fori_loop(0, j - i, lambda t, c: f(r + t * dr, g, at + t * da, c), carry)
                i = j
            return carry

        def prepare(pc, hs):
            if not pc.coded:
                if pc.phase < 2:
                    for h in hs:
                        put(sbuf, h, pc.slot, get(wbuf, h, pc.row // 4, pc.rows // 4))
                return
            emax, gmax = {}, {}
            for h in hs:
                ms = get(mbuf, h, pc.row // 16, pc.rows // 16)
                while len(ms) > 1:
                    ms = [jnp.maximum(*ms[j:j + 2]) if j + 1 < len(ms) else ms[j] for j in range(0, len(ms), 2)]
                emax[h] = jnp.maximum(srl(ms[0], I32(23)), 7)
                g = jnp.max(jnp.max(emax[h].astype(jnp.float32), axis=1, keepdims=True), axis=0, keepdims=True)
                gmax[h] = jnp.broadcast_to(g, (8, 128)).astype(I32)

            def enc(r, g, at, st):
                new = []
                for h, z in zip(hs, st):
                    ps, z = _encode_group(get(wbuf, h, r // 4, g // 4), emax[h] - 7, z)
                    put(sbuf, h, at, ps)
                    new.append(z)
                return tuple(new)
            st = over_groups(pc.groups[::-1], enc, ((_splat(0),) * 4,) * len(hs))
            fin = [_encode_finish(gmax[h], emax[h], z) for h, z in zip(hs, st)]
            for h, (side, over) in zip(hs, fin):
                sbuf[h, pc.slot] = side
                spilled[2 * pc.sem + h] = over.astype(I32)
            for h, (side, over) in zip(hs, fin):
                @pl.when(over)
                def _():
                    sbuf[h, pc.slot] = _splat(0xFFFFFFFF)

                    @pl.loop(0, pc.rows // 4)
                    def _(j):
                        sbuf[h, pc.slot + 1 + j] = wbuf[h, pc.row // 4 + j]

        def start(pc, h):
            for k in range(len(pc.cuts)):
                copy(pc, h, k).start()
            if pc.coded:
                @pl.when(spilled[2 * pc.sem + h] != 0)
                def _():
                    copy(pc, h, len(pc.cuts)).start()

        def finish(pc, h):
            for k in range(len(pc.cuts)):
                copy(pc, h, k).wait_send()
            if pc.coded:
                @pl.when(spilled[2 * pc.sem + h] != 0)
                def _():
                    copy(pc, h, len(pc.cuts)).wait_send()

        def recv(pc, hs, use, before_last=lambda: None):
            done = 0
            for k, (_, _, upto) in enumerate(pc.cuts):
                if k == len(pc.cuts) - 1:
                    before_last()
                with _scope(f"w{pc.phase}.{pc.row}"):
                    for h in hs:
                        copy(pc, h, k).wait_recv()
                if not pc.coded:
                    if pc.phase < 2:
                        for h in hs:
                            use(h, pc.row, 0, _from_words(get(rbuf, half[h], pc.slot, pc.rows // 4)))
                    return
                if k == 0:
                    head = {h: rbuf[half[h], pc.slot, 0, 0] for h in hs}
                    init = [_decode_start(rbuf[half[h], pc.slot], head[h]) for h in hs]
                    st = tuple(z for _, z in init)

                def dec(r, g, at, st):
                    new = []
                    for h, (b2, _), z in zip(hs, init, st):
                        ws, z = _decode_group(get(rbuf, half[h], at, _packed(g // 4)), g // 4, b2, z)
                        use(h, pc.row, r - pc.row, _from_words(ws))
                        new.append(z)
                    return tuple(new)
                st = over_groups(pc.groups[done:upto], dec, st)
                done = upto
            for h in hs:
                @pl.when(head[h] < 0)
                def _():
                    copy(pc, h, len(pc.cuts)).wait_recv()

                    @pl.loop(0, pc.rows // 16)
                    def _(j):
                        use(h, pc.row, j * 16, _from_words(get(rbuf, half[h], pc.slot + 1 + j * 4, 4)))

        def local(r0, dr, n):
            r = r0 + dr
            return r, pl.ds(r if isinstance(r, int) else pl.multiple_of(r, 16), n)

        def out_rows(base, h, r0, dr, n):
            return pl.ds(pl.multiple_of((xrow[h] - C if r0 >= C else base[h]) + r0 + dr, 16), n)

        def use1(h, r0, dr, v):
            r, sl = local(r0, dr, v.shape[0])
            t = xk[h, sl] + v.astype(jnp.float32)
            part[h, sl] = t
            stage(h, r, t)

        def use2(h, r0, dr, v):
            r, sl = local(r0, dr, v.shape[0])
            t = (part[h, sl] + v.astype(jnp.float32)).astype(jnp.bfloat16)
            o_ref[out_rows(keep, h, r0, dr, v.shape[0])] = t
            stage(h, r, t)

        def use3(h, r0, dr, v):
            o_ref[out_rows(give, h, r0, dr, v.shape[0])] = v

        def when_bit(b, f):
            for h in range(2 * (EXTRA > 0)):
                pl.when(bit[h] == b)(lambda: f(h))

        def send_extra(s):
            def f(h):
                if s == 0:
                    stage(h, C, xk[h, pl.ds(C, EXTRA)])
                else:
                    recv(extra[s - 1], (h,), (use1, use2)[s - 1])
                prepare(extra[s], (h,))
                start(extra[s], h)
            when_bit(int(s > 0), f)

        for i, pc in enumerate(phs[0]):
            if i == KEEP_AT:
                for d in ldk:
                    d.start()
            with _scope(f"s0.{pc.row}"):
                for hs in ((0,), (1,)) if i in SOLO or not pc.coded else ((0, 1),):
                    for h in hs:
                        lds[h, i].wait()
                        stage(h, pc.row, xs[h, pl.ds(pc.row, pc.rows)])
                    prepare(pc, hs)
                    if 0 in hs:
                        start(pc, 0)
                if i > LATE:
                    start(pc, 1)
                else:
                    pl.when(odd == 0)(lambda: start(pc, 1))
                if i == LATE:
                    @pl.when(odd == 1)
                    def _():
                        pl.semaphore_wait(ready, 1)
                        for q in phs[0][:i + 1]:
                            start(q, 1)
        for d in ldk:
            d.wait()
        send_extra(0)

        for s, use in ((1, use1), (2, use2)):
            k = 0
            for i, pc in enumerate(phs[s]):
                if i == XAT[s]:
                    send_extra(s)
                while k < len(phs[s - 1]) and phs[s - 1][k].row < pc.row + pc.rows:
                    recv(phs[s - 1][k], (0, 1), use)
                    k += 1
                with _scope(f"s{s}.{pc.row}"):
                    prepare(pc, (0, 1))
                    for h in range(2):
                        start(pc, h)
            if XAT[s] >= len(phs[s]):
                send_extra(s)

        def drain():
            for s in range(3):
                when_bit(int(s > 0), lambda h: finish(extra[s], h))
            for pc in phs[0] + phs[1] + phs[2]:
                for h in range(2):
                    finish(pc, h)

        for i, pc in enumerate(phs[2]):
            if i == XAT[2]:
                when_bit(0, lambda h: recv(extra[2], (h,), use3))
            recv(pc, (0, 1), use3, drain if pc is phs[2][-1] else lambda: None)

    f32 = pltpu.VMEM((2, R, N), jnp.float32)
    words = lambda n: pltpu.VMEM((2, n, 8, 128), I32)
    sem = lambda n: pltpu.SemaphoreType.DMA((2 * n,))
    return pl.pallas_call(
        body,
        out_shape=pltpu.VMEM((M, N), jnp.bfloat16),
        in_specs=[pl.BlockSpec(memory_space=pltpu.HBM)],
        out_specs=pl.BlockSpec(memory_space=pltpu.VMEM),
        scratch_shapes=[f32, f32, f32, words(R // 4), words(R // 16), words(nslot), words(nslot),
                        pltpu.SMEM((2 * nsem,), I32), sem(n1 + 2), sem(nsem), sem(nsem),
                        pltpu.SemaphoreType.REGULAR],
        compiler_params=pltpu.CompilerParams(collective_id=0, **CP),
    )(x)
```

```python
import jax
import jax.numpy as jnp
from jax import lax
from jax.experimental import pallas as pl
from jax.experimental.pallas import tpu as pltpu

M, N = 2048, 512
Q = M // 4
B = Q // 2
GROUPS = B // 32
STEP = 4

CUTS = (
    (16, 16, 32, 48, 64, 48, 32),
    (128, 128),
    (64, 128, 64),
    (128, 128),
    (128, 128),
    (64, 96, 64, 32),
)
FRONT = (7, 1, 2, 1, 1, 1)
LATE = 3
ROUND = 32

POOL = (0, 9, 10, 11)
LEVELS = ((0, 11), (11, 1), (12, 21))
RUN = 6
HEADER = 13

I32 = jnp.int32
srl, sll = lax.shift_right_logical, lax.shift_left
VREGS = (2, 8, 128)


def _i(v):
    return I32(v - (1 << 32) if v >= (1 << 31) else v)


def _splat(v):
    return jnp.full(VREGS, _i(v), I32)


def _sublane():
    return lax.broadcasted_iota(I32, VREGS, 1)


def _header_bits():
    lane = lax.broadcasted_iota(I32, VREGS, 2)
    return jnp.where((_sublane() == 0) & (lane == 0), HEADER, 0)


def _row(v, s):
    return jnp.broadcast_to(v[:, s : s + 1], VREGS)


def _both(v):
    return sll(v, I32(16)) | v


def _running_sum(v):
    for d in (1, 2, 4):
        v = v + jnp.where(_sublane() >= d, pltpu.roll(v, d, 1), 0)
    return v


def _rotate(v, n, up):
    for d in (1, 2, 4):
        v = jnp.where((n & d) != 0, pltpu.roll(v, 8 - d if up else d, 1), v)
    return v


def _shift_right(ws, n):
    rest = [srl(w, n) | sll(sll(u, I32(1)), n ^ 31) for u, w in zip(ws, ws[1:])]
    return [srl(ws[0], n)] + rest


def _shift_left(ws, n):
    rest = [sll(w, n) | srl(srl(u, I32(1)), n ^ 31) for w, u in zip(ws, ws[1:])]
    return rest + [sll(ws[-1], n)]


def _split(v):
    w = pltpu.bitcast(v.astype(jnp.bfloat16), I32)
    a, b = w[..., : N // 2], w[..., N // 2 :]
    rest = sll(b & _i(0x007F007F), I32(7)) | srl(b & _i(0x80008000), I32(1))
    return w & _i(0x7F807F80), (a & _i(0x807F807F)) | rest


def _join(e, m):
    b = (srl(m, I32(7)) & _i(0x007F007F)) | (sll(m, I32(1)) & _i(0x80008000))
    w = jnp.concatenate([m & _i(0x807F807F), b], axis=-1) | e
    return pltpu.bitcast(w, jnp.bfloat16)


def _pick_window(sample):
    t = sum(sample[..., j : j + 128] for j in range(0, N, 128))
    t = (srl(t, I32(16)) + (t & 0xFFFF)).astype(jnp.float32)
    t = jnp.sum(jnp.sum(t, axis=2, keepdims=True), axis=1, keepdims=True)
    mean = jnp.broadcast_to(t, VREGS) * (1.0 / (16 * N)) + 0.12
    whole = mean.astype(I32)
    rank = (7.9 - 6.3 * (mean - whole.astype(jnp.float32))).astype(I32)
    return jnp.clip(whole - 1, 0, 251), jnp.clip(rank, 1, 7)


def _encode_group(es, window, state):
    base, rank, above = window
    string, total, bad = state
    guard, top = _i(0x80008000), _splat(1 << 31)
    fence_lo, fence_hi = _both(base) | guard, guard - _both(base + 4)
    rank2, skip2, above2 = _both(rank), _both(rank - 1), _both(above)
    hi, lo = top, _splat(0)
    size = codes = _splat(0)
    for i in reversed(range(8)):
        e = es[:, i // 4 * 8 : i // 4 * 8 + 8, i % 4 * 128 : i % 4 * 128 + 128]
        t = fence_lo - e
        g = t & guard
        one = srl(g, I32(15))
        low = g - one
        g = (t - skip2) & guard
        skip = above2 & (g - srl(g, I32(15)))
        u = e + fence_hi
        g = u & guard
        high = g - srl(g, I32(15))
        n = (t & low) + one + skip + ((u + rank2) & high)
        codes = codes | sll(t & _i(0x00030003) & ~(low | high), I32(2 * i))
        n_hi = srl(n, I32(16))
        n = n_hi + (n & 0xFFFF)
        size, bad = size + n, bad | n
        lo = srl(lo, n) | sll(hi, n ^ 31)
        hi = srl(hi, n) | top | srl(top, n_hi)
    far = size >= 32
    string = [jnp.where(far, u, w) for u, w in zip([0] + string, string)]
    string = _shift_right(string, size & 31)
    string[0], string[1] = string[0] | hi, string[1] | sll(lo, I32(1))
    bad = bad | srl(size + 1, I32(1))
    return codes, (string, total + size, bad)


def _encode_finish(window, state, tmp):
    base, rank, above = window
    string, total, bad = state
    total = total + above
    bad = (srl(bad | above, I32(5)) != 0) | (total > 32 * RUN)
    string = _shift_right(string, (above - 1) & 31)
    end = _running_sum(total + _header_bits())
    start = end - total
    string = _shift_right(string + [_splat(0)], start & 31) + [_splat(0)] * (7 - RUN)
    for j, w in enumerate(string):
        tmp[:, pl.ds(8 * j, 8)] = w
    first = srl(start, I32(5))
    pool = [_splat(0)] * len(POOL)
    for s in range(8):
        q = _row(first, s)
        w = _rotate(tmp[:, pl.ds(s, 8, stride=8)], q, up=False)
        at = srl(q + ((_sublane() - q) & 7), I32(3))
        pool = [v | jnp.where(at == j, w, 0) for j, v in enumerate(pool)]
    need = jnp.where(bad, 2000, end).astype(jnp.float32)
    need = [jnp.max(need[h]) for h in range(2)]
    level = [(v > 3 * 256).astype(I32) + (v > 4 * 256).astype(I32) for v in need]
    header = sll(base, I32(22)) | sll(rank, I32(19))
    pool[0] = pool[0] | jnp.where(_header_bits() != 0, header, 0)
    return pool, level


def _decode_start(codes, pool, header, tmp):
    ones = _splat(1)
    for v in codes:
        ones = ones + lax.population_count(~(v | srl(v, I32(1))) & _i(0x55555555))
    before = _running_sum(ones) - ones
    pool = [srl(sll(pool[0], _header_bits()), _header_bits())] + pool[1:]
    first = passed = upto = _splat(0)
    for v in pool:
        seen = _running_sum(lax.population_count(v)) + upto
        for s in range(8):
            upto = _row(seen, s)
            ok = upto < before
            first, passed = jnp.where(ok, first + 1, first), jnp.where(ok, upto, passed)
    for s in range(8):
        q = _row(first, s)
        at = srl(q + ((_sublane() - q) & 7), I32(3))
        w = _splat(0)
        for j, v in enumerate(pool):
            w = jnp.where(at == j, v, w)
        tmp[:, pl.ds(8 * s, 8)] = _rotate(w, q, up=True)
    string = [tmp[:, pl.ds(j, 8, stride=8)] for j in range(RUN + 2)]
    left, w, skip = before - passed, string[0], _splat(0)
    for d in (16, 8, 4, 2, 1):
        c = lax.population_count(srl(w, I32(32 - d)))
        ok = c < left
        left, skip = jnp.where(ok, left - c, left), jnp.where(ok, skip + d, skip)
        w = jnp.where(ok, sll(w, I32(d)), w)
    opening = _sublane() == 0
    string = _shift_left(string, jnp.where(opening, _header_bits(), skip))[: RUN + 1]
    lead = lax.clz(jnp.where(opening, string[0], string[0] & _i(0x7FFFFFFF)) | 1)
    above = jnp.where(opening, lead + 1, lead)
    base, rank = srl(header, I32(22)) & 255, srl(header, I32(19)) & 7
    return (base, rank, above), _shift_left(string, lead)[:RUN]


def _decode_group(codes, window, string):
    base, rank, above = window
    roof = sll(_both(base + 4), I32(7))
    hi, lo = string[0], sll(string[0], I32(31)) | srl(string[1], I32(1))
    size, es = _splat(0), []
    for i in range(8):
        e, took = roof, []
        for at, to in ((16 + 2 * i, 23), (2 * i, 7)):
            code = srl(codes, I32(at)) & 3
            n = lax.clz(hi & _i(0x7FFFFFFF))
            u = rank - n
            drop = jnp.where(u > -above, jnp.where(u > 0, n + 3, u), n + (3 - above))
            e = e - sll(jnp.where(code == 0, drop, code), I32(to))
            took.append(jnp.where(code == 0, n, 0))
            hi = sll(hi, took[-1])
        n = took[0] + took[1]
        hi, lo = hi | srl(lo, n ^ 31), sll(lo, n)
        size = size + n
        es.append(e)
    far = size >= 32
    string = [jnp.where(far, u, w) for w, u in zip(string, string[1:] + [0])]
    es = [jnp.concatenate(es[i : i + 4], axis=2) for i in (0, 4)]
    return jnp.concatenate(es, axis=1), _shift_left(string, size & 31)


def _rows(r, n, unit=16):
    return pl.ds(r if isinstance(r, int) else pl.multiple_of(r, unit), n)


def _pairs(r, n):
    return _rows(r // 2, n // 2, 8)


def pallas_dist_ar_i_i_m2048_n512_kernel(x: jax.Array):
    cuts = [[(sum(c[:k]), n) for k, n in enumerate(c)] for c in CUTS]
    sem0 = [sum(len(c) + len(LEVELS) for c in CUTS[:b]) for b in range(7)]

    def body(x_hbm, out, x_give, x_keep, x_far, via, exps, peaks, decoded, tmp,
             bytes_out, bytes_in, exps_out, exps_in, levels, ld, snd, rcv, ready):
        p = lax.axis_index("i")
        odd = p & 1
        half = [(p == 3).astype(I32) ^ h for h in range(2)]
        nbr = [p ^ (1 + 2 * v) for v in half]
        bit = [jnp.where(v == 0, (p ^ (p >> 1)) & 1, p >> 1) for v in half]
        keep = [(2 * half[h] + bit[h]) * Q for h in range(2)]
        give = [(2 * half[h] + 1 - bit[h]) * Q for h in range(2)]

        def signal(sem):
            for to in nbr:
                pl.semaphore_signal(sem, 1, device_id=(to,), device_id_type=pl.DeviceIdType.MESH)

        def load(dst, base, k, r, n):
            return [
                pltpu.make_async_copy(
                    x_hbm.at[_rows(base[h] + r, n)], dst.at[h, pl.ds(r, n)], ld.at[2 * k + h])
                for h in range(2)
            ]

        def remote(src, dst, k, h, to, incoming):
            there = h if incoming else half[h] ^ (to == 3).astype(I32)
            return pltpu.make_async_remote_copy(
                src, dst(there), snd.at[2 * k + h], rcv.at[2 * k + there],
                device_id=(to,), device_id_type=pl.DeviceIdType.MESH)

        def block_copy(src, dst, b, h, part, k, incoming):
            return remote(src.at[b, h, part], lambda j: dst.at[b, j, part], sem0[b] + k,
                          h, nbr[h ^ (b // 2 == 1)], incoming)

        def exp_copy(b, h, level, incoming=False):
            return block_copy(exps_out, exps_in, b, h, pl.ds(*LEVELS[level]), level, incoming)

        def with_byte_copy(b, h, k, act, incoming=False):
            def copy(omit):
                part = _pairs(cuts[b][k][0], cuts[b][k][1] - omit)
                return block_copy(bytes_out, bytes_in, b, h, part, len(LEVELS) + k, incoming)

            if (b, k) == (1, len(cuts[1]) - 1):
                short = p == 0 if incoming else odd > h
                pl.when(short)(lambda: act(copy(ROUND)))
                pl.when(~short)(lambda: act(copy(0)))
            else:
                act(copy(0))

        def detour(h, incoming=False):
            return remote(via.at[2], lambda j: via.at[j], sem0[6], h, 2 + 0 * p, incoming)

        def send_bytes(b, h, k):
            with_byte_copy(b, h, k, lambda d: d.start())

        def wait_bytes(b, ks):
            for k in ks:
                for h in range(2):
                    with_byte_copy(b, h, k, lambda d: d.wait_recv(), incoming=True)

        def stage(b, hs, r, v):
            n = v.shape[1]
            e, m = _split(v)
            bytes_out[b, hs, _pairs(r, n)] = m
            exps[hs, _pairs(r, n)] = srl(e, I32(7))
            hi, lo = (lax.bitcast_convert_type(u, jnp.float32) for u in (e, sll(e, I32(16))))
            t = jnp.maximum(hi, lo)
            t = jnp.maximum(t[..., :256], t[..., 256:])
            peaks[hs, _pairs(r, n)] = jnp.maximum(t[..., :128], t[..., 128:])

        def each_64_rows(f, then_send=None):
            @pl.loop(0, B // 64)
            def _(t):
                f(t * 64)
                for k in range(FRONT[then_send] if then_send else 0):
                    @pl.when(t == sum(cuts[then_send][k]) // 64 - 1)
                    def _():
                        for h in range(2):
                            send_bytes(then_send, h, k)

        def encode_and_send(b, base, rank):
            t, n = peaks[...], B // 2
            while n > 8:
                n //= 2
                t = jnp.maximum(t[:, :n], t[:, n:])
            top = srl(lax.bitcast_convert_type(t, I32), I32(23)) & 255
            window = (base, rank, jnp.where(top > base + 4, top - base - 3, 1))

            def step(t, state):
                for k in range(STEP):
                    g = GROUPS - 1 - k - STEP * t
                    exps_out[b, :, 1 + g], state = _encode_group(
                        exps[:, _pairs(32 * g, 32)], window, state)
                return state

            state = ([_splat(0)] * RUN, _splat(0), _splat(0))
            pool, level = _encode_finish(window, lax.fori_loop(0, GROUPS // STEP, step, state), tmp)
            for at, v in zip(POOL[1:], pool[1:]):
                exps_out[b, :, at] = v
            for h in range(2):
                corner = jnp.where(_header_bits()[h] != 0, sll(level[h], I32(30)), 0)
                exps_out[b, h, 0] = pool[0][h] | corner
                levels[2 * b + h] = level[h]

                @pl.when(level[h] == 2)
                def _():
                    exps_out[b, h, 0] = corner

                    @pl.loop(0, B // 16)
                    def _(j):
                        e = exps[h, _pairs(16 * j, 16)]
                        e = e[:, :256] | sll(e[:, 256:], I32(8))
                        exps_out[b, h, 1 + 2 * j] = e[:, :128]
                        exps_out[b, h, 2 + 2 * j] = e[:, 128:]

                exp_copy(b, h, 0).start()
                for k in (1, 2):
                    pl.when(level[h] >= k)(lambda: exp_copy(b, h, k).start())
                for k in range(FRONT[b], len(cuts[b])):
                    send_bytes(b, h, k)

        def wait_and_decode(b):
            for h in range(2):
                exp_copy(b, h, 0, incoming=True).wait_recv()
            header = [exps_in[b, h, 0, 0, 0] for h in range(2)]
            level = [srl(v, I32(30)) for v in header]
            for h in range(2):
                @pl.when(level[h] == 0)
                def _():
                    exps_in[b, h, POOL[-1]] = jnp.zeros((8, 128), I32)

                for k in (1, 2):
                    pl.when(level[h] >= k)(lambda: exp_copy(b, h, k, incoming=True).wait_recv())

            @pl.when((level[0] < 2) | (level[1] < 2))
            def _():
                use = [jnp.where(level[h] < 2, h, 1 - h) for h in range(2)]
                head = [jnp.where(level[h] < 2, header[h], header[1 - h]) for h in range(2)]
                vreg = lambda at: jnp.stack([exps_in[b, use[h], at] for h in range(2)])
                window, string = _decode_start(
                    [vreg(1 + g) for g in range(GROUPS)], [vreg(at) for at in POOL],
                    jnp.stack([jnp.full((8, 128), v, I32) for v in head]), tmp)

                def step(t, string):
                    for k in range(STEP):
                        g = STEP * t + k
                        decoded[:, _pairs(32 * g, 32)], string = _decode_group(
                            vreg(1 + g), window, string)
                    return string

                lax.fori_loop(0, GROUPS // STEP, step, string)

            for h in range(2):
                @pl.when(level[h] == 2)
                def _():
                    @pl.loop(0, B // 16)
                    def _(j):
                        v = [exps_in[b, h, k + 2 * j] for k in (1, 2)]
                        v = [sll(u, I32(7)) for u in v] + [srl(u, I32(1)) for u in v]
                        decoded[h, _pairs(16 * j, 16)] = jnp.concatenate(v, axis=1) & _i(0x7F807F80)

        def received(b, r, n):
            return _join(decoded[:, _pairs(r, n)], bytes_in[b, :, _pairs(r, n)])

        def write(base, r, v):
            for h in range(2):
                out[_rows(base[h] + r, v.shape[1])] = v[h]

        def wait_sent(b):
            for h in range(2):
                for k in range(len(cuts[b])):
                    with_byte_copy(b, h, k, lambda d: d.wait_send())
                exp_copy(b, h, 0).wait_send()
                for k in (1, 2):
                    pl.when(levels[2 * b + h] >= k)(lambda: exp_copy(b, h, k).wait_send())

        give_loads = [load(x_give, give, k, r, n) for k, (r, n) in enumerate(cuts[0] + [(B, B)])]
        keep_loads = [load(x_keep, keep, len(give_loads) + k, k * B, B) for k in range(2)]
        far_load = pltpu.make_async_copy(
            x_hbm.at[_rows(give[0] + Q - ROUND, ROUND)], x_far, ld.at[2 * len(give_loads) + 4])

        give_loads[0][0].start()
        barrier = pltpu.get_barrier_semaphore()
        pl.when(p != 2)(lambda: signal(barrier))

        @pl.when(p == 2)
        def _():
            pl.semaphore_wait(barrier, 2)
            signal(ready)

        early = sum(give_loads[:-1], [])
        early.insert(2 * LATE + 2, far_load)
        for d in early[1:]:
            d.start()
        pl.when(p == 0)(lambda: pl.semaphore_wait(barrier, 2))
        pl.when(odd == 1)(lambda: pl.semaphore_wait(barrier, 1))

        for k, (r, n) in enumerate(cuts[0]):
            for h in range(2):
                give_loads[k][h].wait()
                stage(0, pl.ds(h, 1), r, x_give[pl.ds(h, 1), pl.ds(r, n)])
                if h == 0 or k >= LATE:
                    send_bytes(0, h, k)
                else:
                    pl.when(odd == 0)(lambda: send_bytes(0, 1, k))
                if k == 0:
                    give_loads[-1][h].start()
                if (k, h) == (LATE, 0):
                    base, rank = _pick_window(exps[:, :8])

                    @pl.when(odd == 1)
                    def _():
                        pl.semaphore_wait(ready, 1)
                        for j in range(LATE):
                            send_bytes(0, 1, j)

                if (k, h) == (LATE, 1):
                    far_load.wait()

                    @pl.when(odd == 1)
                    def _():
                        via[2] = x_far[...].astype(jnp.bfloat16)
                        detour(0).start()

        for d in keep_loads[0]:
            d.start()
        encode_and_send(0, base, rank)
        for d in keep_loads[1]:
            d.start()
        for d in give_loads[-1]:
            d.wait()
        both = slice(None)
        each_64_rows(lambda r: stage(1, both, r, x_give[:, _rows(B + r, 64)]), then_send=1)

        @pl.when(p == 2)
        def _():
            for h in range(2):
                detour(h, incoming=True).wait_recv()
            t = x_give[:, pl.ds(Q - ROUND, ROUND)] + via[:2].astype(jnp.float32)
            stage(1, both, B - ROUND, t)

        encode_and_send(1, *_pick_window(exps[:, :8]))

        for b in range(4):
            r0 = b % 2 * B
            wait_and_decode(b)
            wait_bytes(b, range(len(cuts[b])))
            if b < 2:
                for d in keep_loads[b]:
                    d.wait()
            if b == 1:
                @pl.when(p == 0)
                def _():
                    gone = _pairs(B - ROUND, ROUND)
                    bytes_in[1, :, gone] = jnp.zeros((2, ROUND // 2, N // 2), I32)
                    decoded[:, gone] = jnp.zeros((2, ROUND // 2, N), I32)

            def add(r):
                t = x_keep[:, _rows(r0 + r, 64)] + received(b, r, 64).astype(jnp.float32)
                if b < 2:
                    x_keep[:, _rows(r0 + r, 64)] = t
                else:
                    write(keep, r0 + r, t.astype(jnp.bfloat16))
                stage(b + 2, both, r, t)

            each_64_rows(add, then_send=b + 2)
            encode_and_send(b + 2, *_pick_window(exps[:, :8]))

        wait_and_decode(4)
        wait_bytes(4, range(len(cuts[4])))
        each_64_rows(lambda r: write(give, r, received(4, r, 64)))
        for b in range(5):
            wait_sent(b)
        pl.when(odd == 1)(lambda: detour(0).wait_send())
        wait_and_decode(5)
        for k, (r, n) in enumerate(cuts[5]):
            if k == len(cuts[5]) - 1:
                wait_sent(5)
            wait_bytes(5, [k])
            write(give, B + r, received(5, r, n))

    f32, vmem, dma = jnp.float32, pltpu.VMEM, pltpu.SemaphoreType.DMA
    return pl.pallas_call(
        body,
        out_shape=vmem((M, N), jnp.bfloat16),
        in_specs=[pl.BlockSpec(memory_space=pltpu.HBM)],
        out_specs=pl.BlockSpec(memory_space=vmem),
        scratch_shapes=[
            vmem((2, Q, N), f32),
            vmem((2, Q, N), f32),
            vmem((ROUND, N), f32),
            vmem((3, ROUND, N), jnp.bfloat16),
            vmem((2, B // 2, N), I32),
            vmem((2, B // 2, 128), f32),
            vmem((2, B // 2, N), I32),
            vmem((2, 72, 128), I32),
            vmem((6, 2, B // 2, N // 2), I32),
            vmem((6, 2, B // 2, N // 2), I32),
            vmem((6, 2, sum(LEVELS[-1]), 8, 128), I32),
            vmem((6, 2, sum(LEVELS[-1]), 8, 128), I32),
            pltpu.SMEM((12,), I32),
            dma((2 * len(CUTS[0]) + 8,)),
            dma((2 * sem0[6] + 2,)),
            dma((2 * sem0[6] + 2,)),
            pltpu.SemaphoreType.REGULAR,
        ],
        compiler_params=pltpu.CompilerParams(collective_id=0, disable_semaphore_checks=True),
    )(x)
```

```python
import jax
import jax.numpy as jnp
from jax import lax
from jax.experimental import pallas as pl
from jax.experimental.pallas import tpu as pltpu

M, N = 2048, 512
Q = M // 4
B = Q // 2
GROUPS = B // 32
STEP = 8

CUTS = (
    (16, 16, 32, 48, 64, 48, 32),
    (128, 128),
    (64, 128, 64),
    (128, 128),
    (128, 128),
    (64, 96, 64, 16, 16),
)
FRONT = (7, 1, 2, 1, 1, 1)
LATE = 3
ROUND = 32

POOL = (8, 9, 10, 11)
LEVELS = ((0, 11), (11, 1), (12, 22))
RUN = 6
HEADER = 13

I32 = jnp.int32
srl, sll = lax.shift_right_logical, lax.shift_left
VREGS = (2, 8, 128)


def _i(v):
    return I32(v - (1 << 32) if v >= (1 << 31) else v)


def _splat(v):
    return jnp.full(VREGS, _i(v), I32)


def _sublane():
    return lax.broadcasted_iota(I32, VREGS, 1)


def _header_bits():
    lane = lax.broadcasted_iota(I32, VREGS, 2)
    return jnp.where((_sublane() == 0) & (lane == 0), HEADER, 0)


def _row(v, s):
    return jnp.broadcast_to(v[:, s : s + 1], VREGS)


def _both(v):
    return sll(v, I32(16)) | v


def _running_sum(v):
    for d in (1, 2, 4):
        v = v + jnp.where(_sublane() >= d, pltpu.roll(v, d, 1), 0)
    return v


def _rotate(v, n, up):
    for d in (1, 2, 4):
        v = jnp.where((n & d) != 0, pltpu.roll(v, 8 - d if up else d, 1), v)
    return v


def _shift_right(ws, n):
    rest = [srl(w, n) | sll(sll(u, I32(1)), n ^ 31) for u, w in zip(ws, ws[1:])]
    return [srl(ws[0], n)] + rest


def _shift_left(ws, n):
    rest = [sll(w, n) | srl(srl(u, I32(1)), n ^ 31) for w, u in zip(ws, ws[1:])]
    return rest + [sll(ws[-1], n)]


def _split(v):
    w = pltpu.bitcast(v.astype(jnp.bfloat16), I32)
    a, b = w[..., : N // 2], w[..., N // 2 :]
    rest = sll(b & _i(0x007F007F), I32(7)) | srl(b & _i(0x80008000), I32(1))
    return w & _i(0x7F807F80), (a & _i(0x807F807F)) | rest


def _join(e, m):
    b = (srl(m, I32(7)) & _i(0x007F007F)) | (sll(m, I32(1)) & _i(0x80008000))
    w = jnp.concatenate([m & _i(0x807F807F), b], axis=-1) | e
    return pltpu.bitcast(w, jnp.bfloat16)


def _pick_window(sample):
    t = sum(sample[..., j : j + 128] for j in range(0, N, 128))
    t = (srl(t, I32(16)) + (t & 0xFFFF)).astype(jnp.float32)
    t = jnp.sum(jnp.sum(t, axis=2, keepdims=True), axis=1, keepdims=True)
    mean = jnp.broadcast_to(t, VREGS) * (1.0 / (16 * N)) + 0.12
    whole = mean.astype(I32)
    rank = (7.9 - 6.3 * (mean - whole.astype(jnp.float32))).astype(I32)
    return jnp.clip(whole - 1, 0, 251), jnp.clip(rank, 1, 7)


def _encode_group(es, window, state):
    base, rank, above = window
    string, total, bad = state
    guard, top = _i(0x80008000), _splat(1 << 31)
    fence_lo, fence_hi = _both(base) | guard, guard - _both(base + 4)
    rank2, skip2, above2 = _both(rank), _both(rank - 1), _both(above)
    hi, lo = top, _splat(0)
    size = codes = _splat(0)
    for i in reversed(range(8)):
        e = es[:, i // 4 * 8 : i // 4 * 8 + 8, i % 4 * 128 : i % 4 * 128 + 128]
        t = fence_lo - e
        g = t & guard
        one = srl(g, I32(15))
        low = g - one
        g = (t - skip2) & guard
        skip = above2 & (g - srl(g, I32(15)))
        u = e + fence_hi
        g = u & guard
        high = g - srl(g, I32(15))
        n = (t & low) + one + skip + ((u + rank2) & high)
        codes = codes | sll(t & _i(0x00030003) & ~(low | high), I32(2 * i))
        n_hi = srl(n, I32(16))
        n = n_hi + (n & 0xFFFF)
        size, bad = size + n, bad | n
        lo = srl(lo, n) | sll(hi, n ^ 31)
        hi = srl(hi, n) | top | srl(top, n_hi)
    far = size >= 32
    string = [jnp.where(far, u, w) for u, w in zip([0] + string, string)]
    string = _shift_right(string, size & 31)
    string[0], string[1] = string[0] | hi, string[1] | sll(lo, I32(1))
    bad = bad | srl(size + 1, I32(1))
    return codes, (string, total + size, bad)


def _encode_finish(window, state, tmp):
    base, rank, above = window
    string, total, bad = state
    total = total + above
    bad = (srl(bad | above, I32(5)) != 0) | (total > 32 * RUN)
    string = _shift_right(string, (above - 1) & 31)
    end = _running_sum(total + _header_bits())
    start = end - total
    string = _shift_right(string + [_splat(0)], start & 31) + [_splat(0)] * (7 - RUN)
    for j, w in enumerate(string):
        tmp[:, pl.ds(8 * j, 8)] = w
    first = srl(start, I32(5))
    pool = [_splat(0)] * len(POOL)
    for s in range(8):
        q = _row(first, s)
        w = _rotate(tmp[:, pl.ds(s, 8, stride=8)], q, up=False)
        at = srl(q + ((_sublane() - q) & 7), I32(3))
        pool = [v | jnp.where(at == j, w, 0) for j, v in enumerate(pool)]
    need = jnp.where(bad, 2000, end).astype(jnp.float32)
    need = [jnp.max(need[h]) for h in range(2)]
    level = [(v > 3 * 256).astype(I32) + (v > 4 * 256).astype(I32) for v in need]
    header = sll(base, I32(22)) | sll(rank, I32(19))
    pool[0] = pool[0] | jnp.where(_header_bits() != 0, header, 0)
    return pool, level


def _decode_start(codes, pool, header, tmp):
    ones = _splat(1)
    for v in codes:
        ones = ones + lax.population_count(~(v | srl(v, I32(1))) & _i(0x55555555))
    before = _running_sum(ones) - ones
    pool = [srl(sll(pool[0], _header_bits()), _header_bits())] + pool[1:]
    first = passed = upto = _splat(0)
    for v in pool:
        seen = _running_sum(lax.population_count(v)) + upto
        for s in range(8):
            upto = _row(seen, s)
            ok = upto < before
            first, passed = jnp.where(ok, first + 1, first), jnp.where(ok, upto, passed)
    for s in range(8):
        q = _row(first, s)
        at = srl(q + ((_sublane() - q) & 7), I32(3))
        w = _splat(0)
        for j, v in enumerate(pool):
            w = jnp.where(at == j, v, w)
        tmp[:, pl.ds(8 * s, 8)] = _rotate(w, q, up=True)
    string = [tmp[:, pl.ds(j, 8, stride=8)] for j in range(RUN + 2)]
    left, w, skip = before - passed, string[0], _splat(0)
    for d in (16, 8, 4, 2, 1):
        c = lax.population_count(srl(w, I32(32 - d)))
        ok = c < left
        left, skip = jnp.where(ok, left - c, left), jnp.where(ok, skip + d, skip)
        w = jnp.where(ok, sll(w, I32(d)), w)
    opening = _sublane() == 0
    string = _shift_left(string, jnp.where(opening, _header_bits(), skip))[: RUN + 1]
    lead = lax.clz(jnp.where(opening, string[0], string[0] & _i(0x7FFFFFFF)) | 1)
    above = jnp.where(opening, lead + 1, lead)
    base, rank = srl(header, I32(22)) & 255, srl(header, I32(19)) & 7
    return (base, rank, above), _shift_left(string, lead)[:RUN]


def _decode_group(codes, window, string):
    base, rank, above = window
    roof = sll(_both(base + 4), I32(7))
    hi, lo = string[0], sll(string[0], I32(31)) | srl(string[1], I32(1))
    size, es = _splat(0), []
    for i in range(8):
        e, took = roof, []
        for at, to in ((16 + 2 * i, 23), (2 * i, 7)):
            code = srl(codes, I32(at)) & 3
            n = lax.clz(hi & _i(0x7FFFFFFF))
            u = rank - n
            drop = jnp.where(u > -above, jnp.where(u > 0, n + 3, u), n + (3 - above))
            e = e - sll(jnp.where(code == 0, drop, code), I32(to))
            took.append(jnp.where(code == 0, n, 0))
            hi = sll(hi, took[-1])
        n = took[0] + took[1]
        hi, lo = hi | srl(lo, n ^ 31), sll(lo, n)
        size = size + n
        es.append(e)
    far = size >= 32
    string = [jnp.where(far, u, w) for w, u in zip(string, string[1:] + [0])]
    es = [jnp.concatenate(es[i : i + 4], axis=2) for i in (0, 4)]
    return jnp.concatenate(es, axis=1), _shift_left(string, size & 31)


def _rows(r, n, unit=16):
    return pl.ds(r if isinstance(r, int) else pl.multiple_of(r, unit), n)


def _pairs(r, n):
    return _rows(r // 2, n // 2, 8)


def _plain_slot(j):
    return j + 1 + (j + 1 >= POOL[0]).astype(I32)


def pallas_dist_ar_i_i_m2048_n512_kernel(x: jax.Array):
    cuts = [[(sum(c[:k]), n) for k, n in enumerate(c)] for c in CUTS]
    sem0 = [sum(len(c) + len(LEVELS) for c in CUTS[:b]) for b in range(7)]

    def body(x_hbm, out, x_give, x_keep, x_far, via, exps, peaks, decoded, tmp,
             bytes_out, bytes_in, exps_out, exps_in, levels, ld, snd, rcv, ready):
        p = lax.axis_index("i")
        odd = p & 1
        half = [(p == 3).astype(I32) ^ h for h in range(2)]
        nbr = [p ^ (1 + 2 * v) for v in half]
        bit = [jnp.where(v == 0, (p ^ (p >> 1)) & 1, p >> 1) for v in half]
        keep = [(2 * half[h] + bit[h]) * Q for h in range(2)]
        give = [(2 * half[h] + 1 - bit[h]) * Q for h in range(2)]

        def signal(sem):
            for to in nbr[::-1]:
                pl.semaphore_signal(sem, 1, device_id=(to,), device_id_type=pl.DeviceIdType.MESH)

        def load(dst, base, k, r, n):
            return [
                pltpu.make_async_copy(
                    x_hbm.at[_rows(base[h] + r, n)], dst.at[h, pl.ds(r, n)], ld.at[2 * k + h])
                for h in range(2)
            ]

        def remote(src, dst, k, h, to, incoming):
            there = h if incoming else half[h] ^ (to == 3).astype(I32)
            return pltpu.make_async_remote_copy(
                src, dst(there), snd.at[2 * k + h], rcv.at[2 * k + there],
                device_id=(to,), device_id_type=pl.DeviceIdType.MESH)

        def block_copy(src, dst, b, h, part, k, incoming):
            return remote(src.at[b, h, part], lambda j: dst.at[b, j, part], sem0[b] + k,
                          h, nbr[h ^ (b // 2 == 1)], incoming)

        def with_copy(copy, act, h, incoming, has_rerouted_rows):
            if has_rerouted_rows:
                short = p == 0 if incoming else odd > h
                pl.when(short)(lambda: act(copy(1)))
                pl.when(~short)(lambda: act(copy(0)))
            else:
                act(copy(0))

        def with_exp_copy(b, h, level, act, incoming=False):
            def copy(omit):
                part = pl.ds(LEVELS[level][0] + omit, LEVELS[level][1] - omit)
                return block_copy(exps_out, exps_in, b, h, part, level, incoming)

            with_copy(copy, act, h, incoming, (b, level) == (1, 0))

        def with_byte_copy(b, h, k, act, incoming=False):
            def copy(omit):
                part = _pairs(cuts[b][k][0], cuts[b][k][1] - omit * ROUND)
                return block_copy(bytes_out, bytes_in, b, h, part, len(LEVELS) + k, incoming)

            with_copy(copy, act, h, incoming, (b, k) == (1, len(cuts[1]) - 1))

        def with_exp_copies(b, h, first, level, act, incoming=False):
            for k in range(first, len(LEVELS)):
                go = lambda: with_exp_copy(b, h, k, act, incoming)
                pl.when(level >= k)(go) if k else go()

        start, sent, landed = (lambda d: d.start()), (lambda d: d.wait_send()), (lambda d: d.wait_recv())

        def detour(h, incoming=False):
            return remote(via.at[2], lambda j: via.at[j], sem0[6], h, 2 + 0 * p, incoming)

        def send_bytes(b, h, k):
            with_byte_copy(b, h, k, start)

        def wait_bytes(b, ks):
            for k in ks:
                for h in range(2):
                    with_byte_copy(b, h, k, landed, incoming=True)

        def stage(b, hs, r, v):
            n = v.shape[1]
            e, m = _split(v)
            bytes_out[b, hs, _pairs(r, n)] = m
            exps[hs, _pairs(r, n)] = srl(e, I32(7))
            hi, lo = (lax.bitcast_convert_type(u, jnp.float32) for u in (e, sll(e, I32(16))))
            t = jnp.maximum(hi, lo)
            t = jnp.maximum(t[..., :256], t[..., 256:])
            peaks[hs, _pairs(r, n)] = jnp.maximum(t[..., :128], t[..., 128:])

        def each_64_rows(f, then_send=None):
            @pl.loop(0, B // 64)
            def _(t):
                f(t * 64)
                for k in range(FRONT[then_send] if then_send else 0):
                    @pl.when(t == sum(cuts[then_send][k]) // 64 - 1)
                    def _():
                        for h in range(2):
                            send_bytes(then_send, h, k)

        def encode_and_send(b, base, rank):
            t, n = peaks[...], B // 2
            while n > 8:
                n //= 2
                t = jnp.maximum(t[:, :n], t[:, n:])
            top = srl(lax.bitcast_convert_type(t, I32), I32(23)) & 255
            window = (base, rank, jnp.where(top > base + 4, top - base - 3, 1))
            if b == 1:
                @pl.when(odd == 1)
                def _():
                    filler = _both(base[0] + 1)
                    exps[0, _pairs(B - ROUND, ROUND)] = jnp.tile(filler, (ROUND // 16, N // 128))

            def step(t, state):
                for k in range(STEP):
                    j = STEP * t + k
                    exps_out[b, :, j], state = _encode_group(
                        exps[:, _pairs(32 * (GROUPS - 1 - j), 32)], window, state)
                return state

            state = ([_splat(0)] * RUN, _splat(0), _splat(0))
            pool, level = _encode_finish(window, lax.fori_loop(0, GROUPS // STEP, step, state), tmp)
            for at, v in zip(POOL[1:], pool[1:]):
                exps_out[b, :, at] = v
            for h in range(2):
                corner = jnp.where(_header_bits()[h] != 0, sll(level[h], I32(30)), 0)
                exps_out[b, h, POOL[0]] = pool[0][h] | corner
                levels[2 * b + h] = level[h]

                @pl.when(level[h] == 2)
                def _():
                    exps_out[b, h, POOL[0]] = corner

                    @pl.loop(0, B // 16)
                    def _(j):
                        e = exps[h, _pairs(16 * j, 16)]
                        e = e[:, :256] | sll(e[:, 256:], I32(8))
                        exps_out[b, h, _plain_slot(2 * j)] = e[:, :128]
                        exps_out[b, h, _plain_slot(2 * j + 1)] = e[:, 128:]

                with_exp_copies(b, h, 0, level[h], start)
                for k in range(FRONT[b], len(cuts[b])):
                    send_bytes(b, h, k)

        def wait_and_decode(b):
            for h in range(2):
                with_exp_copy(b, h, 0, landed, incoming=True)
            if b == 1:
                @pl.when(p == 0)
                def _():
                    exps_in[1, :, 0] = _splat(0xFFFFFFFF)

            header = [exps_in[b, h, POOL[0], 0, 0] for h in range(2)]
            level = [srl(v, I32(30)) for v in header]
            for h in range(2):
                @pl.when(level[h] == 0)
                def _():
                    exps_in[b, h, POOL[-1]] = jnp.zeros((8, 128), I32)

                with_exp_copies(b, h, 1, level[h], landed, incoming=True)

            @pl.when((level[0] < 2) | (level[1] < 2))
            def _():
                use = [jnp.where(level[h] < 2, h, 1 - h) for h in range(2)]
                head = [jnp.where(level[h] < 2, header[h], header[1 - h]) for h in range(2)]
                vreg = lambda at: jnp.stack([exps_in[b, use[h], at] for h in range(2)])
                window, string = _decode_start(
                    [vreg(j) for j in range(GROUPS)], [vreg(at) for at in POOL],
                    jnp.stack([jnp.full((8, 128), v, I32) for v in head]), tmp)

                def step(t, string):
                    for k in range(STEP):
                        g = STEP * t + k
                        decoded[:, _pairs(32 * g, 32)], string = _decode_group(
                            vreg(GROUPS - 1 - g), window, string)
                    return string

                lax.fori_loop(0, GROUPS // STEP, step, string)

            for h in range(2):
                @pl.when(level[h] == 2)
                def _():
                    @pl.loop(0, B // 16)
                    def _(j):
                        v = [exps_in[b, h, _plain_slot(2 * j + k)] for k in range(2)]
                        v = [sll(u, I32(7)) for u in v] + [srl(u, I32(1)) for u in v]
                        decoded[h, _pairs(16 * j, 16)] = jnp.concatenate(v, axis=1) & _i(0x7F807F80)

        def received(b, r, n):
            return _join(decoded[:, _pairs(r, n)], bytes_in[b, :, _pairs(r, n)])

        def write(base, r, v):
            for h in range(2):
                out[_rows(base[h] + r, v.shape[1])] = v[h]

        def wait_sent(b):
            for h in range(2):
                for k in range(len(cuts[b])):
                    with_byte_copy(b, h, k, sent)
                with_exp_copies(b, h, 0, levels[2 * b + h], sent)

        give_loads = [load(x_give, give, k, r, n) for k, (r, n) in enumerate(cuts[0] + [(B, B)])]
        keep_loads = [load(x_keep, keep, len(give_loads) + k, k * B, B) for k in range(2)]
        far_load = pltpu.make_async_copy(
            x_hbm.at[_rows(give[0] + Q - ROUND, ROUND)], x_far, ld.at[2 * len(give_loads) + 4])

        barrier = pltpu.get_barrier_semaphore()
        pl.when(p != 2)(lambda: signal(barrier))
        give_loads[0][0].start()

        @pl.when(p == 2)
        def _():
            pl.semaphore_wait(barrier, 2)
            signal(ready)

        early = sum(give_loads[:-1], [])
        early.insert(2 * LATE + 2, far_load)
        for d in early[1:]:
            d.start()
        pl.when(p == 0)(lambda: pl.semaphore_wait(barrier, 2))
        pl.when(odd == 1)(lambda: pl.semaphore_wait(barrier, 1))

        for k, (r, n) in enumerate(cuts[0]):
            for h in range(2):
                give_loads[k][h].wait()
                stage(0, pl.ds(h, 1), r, x_give[pl.ds(h, 1), pl.ds(r, n)])
                if h == 0 or k >= LATE:
                    send_bytes(0, h, k)
                else:
                    pl.when(odd == 0)(lambda: send_bytes(0, 1, k))
                if k == 0:
                    give_loads[-1][h].start()
                if (k, h) == (LATE, 0):
                    base, rank = _pick_window(exps[:, :8])

                    @pl.when(odd == 1)
                    def _():
                        pl.semaphore_wait(ready, 1)
                        for j in range(LATE):
                            send_bytes(0, 1, j)

                if (k, h) == (LATE, 1):
                    far_load.wait()

                    @pl.when(odd == 1)
                    def _():
                        via[2] = x_far[...].astype(jnp.bfloat16)
                        detour(0).start()

        for d in keep_loads[0]:
            d.start()
        encode_and_send(0, base, rank)
        for d in keep_loads[1]:
            d.start()
        for d in give_loads[-1]:
            d.wait()
        both = slice(None)
        each_64_rows(lambda r: stage(1, both, r, x_give[:, _rows(B + r, 64)]), then_send=1)

        @pl.when(p == 2)
        def _():
            for h in range(2):
                detour(h, incoming=True).wait_recv()
            t = x_give[:, pl.ds(Q - ROUND, ROUND)] + via[:2].astype(jnp.float32)
            stage(1, both, B - ROUND, t)

        encode_and_send(1, *_pick_window(exps[:, :8]))

        for b in range(4):
            r0 = b % 2 * B
            wait_and_decode(b)
            wait_bytes(b, range(len(cuts[b])))
            if b < 2:
                for d in keep_loads[b]:
                    d.wait()
            if b == 1:
                @pl.when(p == 0)
                def _():
                    gone = _pairs(B - ROUND, ROUND)
                    bytes_in[1, :, gone] = jnp.zeros((2, ROUND // 2, N // 2), I32)
                    decoded[:, gone] = jnp.zeros((2, ROUND // 2, N), I32)

            def add(r):
                t = x_keep[:, _rows(r0 + r, 64)] + received(b, r, 64).astype(jnp.float32)
                if b < 2:
                    x_keep[:, _rows(r0 + r, 64)] = t
                else:
                    write(keep, r0 + r, t.astype(jnp.bfloat16))
                stage(b + 2, both, r, t)

            each_64_rows(add, then_send=b + 2)
            encode_and_send(b + 2, *_pick_window(exps[:, :8]))

        wait_and_decode(4)
        wait_bytes(4, range(len(cuts[4])))
        each_64_rows(lambda r: write(give, r, received(4, r, 64)))
        for b in range(5):
            wait_sent(b)
        pl.when(odd == 1)(lambda: detour(0).wait_send())
        wait_and_decode(5)
        for k, (r, n) in enumerate(cuts[5]):
            if k == len(cuts[5]) - 1:
                wait_sent(5)
            wait_bytes(5, [k])
            write(give, B + r, received(5, r, n))

    f32, vmem, dma = jnp.float32, pltpu.VMEM, pltpu.SemaphoreType.DMA
    return pl.pallas_call(
        body,
        out_shape=vmem((M, N), jnp.bfloat16),
        in_specs=[pl.BlockSpec(memory_space=pltpu.HBM)],
        out_specs=pl.BlockSpec(memory_space=vmem),
        scratch_shapes=[
            vmem((2, Q, N), f32),
            vmem((2, Q, N), f32),
            vmem((ROUND, N), f32),
            vmem((3, ROUND, N), jnp.bfloat16),
            vmem((2, B // 2, N), I32),
            vmem((2, B // 2, 128), f32),
            vmem((2, B // 2, N), I32),
            vmem((2, 72, 128), I32),
            vmem((6, 2, B // 2, N // 2), I32),
            vmem((6, 2, B // 2, N // 2), I32),
            vmem((6, 2, sum(LEVELS[-1]), 8, 128), I32),
            vmem((6, 2, sum(LEVELS[-1]), 8, 128), I32),
            pltpu.SMEM((12,), I32),
            dma((2 * len(CUTS[0]) + 8,)),
            dma((2 * sem0[6] + 2,)),
            dma((2 * sem0[6] + 2,)),
            pltpu.SemaphoreType.REGULAR,
        ],
        compiler_params=pltpu.CompilerParams(collective_id=0, disable_semaphore_checks=True),
    )(x)
```

```python
import jax
import jax.numpy as jnp
from jax import lax
from jax.experimental import pallas as pl
from jax.experimental.pallas import tpu as pltpu

M, N = 2048, 512
Q = M // 4
B = Q // 2
GROUPS = B // 32

CUTS = (
    (16, 16, 32, 48, 64, 48, 32),
    (128, 128),
    (64, 128, 64),
    (128, 128),
    (128, 128),
    (64, 96, 64, 16, 16),
)
FRONT = (7, 1, 2, 1, 1, 1)
LATE = 3
ROUND = 32

POOL = (8, 9, 10, 11)
LEVELS = ((0, 11), (11, 1), (12, 22))
RUN = 6
HEADER = 13

I32 = jnp.int32
srl, sll = lax.shift_right_logical, lax.shift_left
VREGS = (2, 8, 128)


def _i(v):
    return I32(v - (1 << 32) if v >= (1 << 31) else v)


def _splat(v):
    return jnp.full(VREGS, _i(v), I32)


def _sublane():
    return lax.broadcasted_iota(I32, VREGS, 1)


def _header_bits():
    lane = lax.broadcasted_iota(I32, VREGS, 2)
    return jnp.where((_sublane() == 0) & (lane == 0), HEADER, 0)


def _row(v, s):
    return jnp.broadcast_to(v[:, s : s + 1], VREGS)


def _both(v):
    return sll(v, I32(16)) | v


def _running_sum(v):
    for d in (1, 2, 4):
        v = v + jnp.where(_sublane() >= d, pltpu.roll(v, d, 1), 0)
    return v


def _rotate(v, n, up):
    for d in (1, 2, 4):
        v = jnp.where((n & d) != 0, pltpu.roll(v, 8 - d if up else d, 1), v)
    return v


def _shift_right(ws, n):
    rest = [srl(w, n) | sll(sll(u, I32(1)), n ^ 31) for u, w in zip(ws, ws[1:])]
    return [srl(ws[0], n)] + rest


def _shift_left(ws, n):
    rest = [sll(w, n) | srl(srl(u, I32(1)), n ^ 31) for w, u in zip(ws, ws[1:])]
    return rest + [sll(ws[-1], n)]


def _split(v):
    w = pltpu.bitcast(v.astype(jnp.bfloat16), I32)
    a, b = w[..., : N // 2], w[..., N // 2 :]
    rest = sll(b & _i(0x007F007F), I32(7)) | srl(b & _i(0x80008000), I32(1))
    return w & _i(0x7F807F80), (a & _i(0x807F807F)) | rest


def _join(e, m):
    b = (srl(m, I32(7)) & _i(0x007F007F)) | (sll(m, I32(1)) & _i(0x80008000))
    w = jnp.concatenate([m & _i(0x807F807F), b], axis=-1) | e
    return pltpu.bitcast(w, jnp.bfloat16)


def _pick_window(sample):
    t = sum(sample[..., j : j + 128] for j in range(0, N, 128))
    t = (srl(t, I32(16)) + (t & 0xFFFF)).astype(jnp.float32)
    t = jnp.sum(jnp.sum(t, axis=2, keepdims=True), axis=1, keepdims=True)
    mean = jnp.broadcast_to(t, VREGS) * (1.0 / (16 * N)) + 0.12
    whole = mean.astype(I32)
    rank = (7.9 - 6.3 * (mean - whole.astype(jnp.float32))).astype(I32)
    return jnp.clip(whole - 1, 0, 251), jnp.clip(rank, 1, 7)


def _encode_group(es, window, state):
    base, rank, above = window
    string, total, bad = state
    guard, top = _i(0x80008000), _splat(1 << 31)
    fence_lo, fence_hi = _both(base) | guard, guard - _both(base + 4)
    rank2, skip2, above2 = _both(rank), _both(rank - 1), _both(above)
    hi, lo = top, _splat(0)
    size = codes = _splat(0)
    for i in reversed(range(8)):
        e = es[:, i // 4 * 8 : i // 4 * 8 + 8, i % 4 * 128 : i % 4 * 128 + 128]
        t = fence_lo - e
        g = t & guard
        one = srl(g, I32(15))
        low = g - one
        g = (t - skip2) & guard
        skip = above2 & (g - srl(g, I32(15)))
        u = e + fence_hi
        g = u & guard
        high = g - srl(g, I32(15))
        n = (t & low) + one + skip + ((u + rank2) & high)
        codes = codes | sll(t & _i(0x00030003) & ~(low | high), I32(2 * i))
        n_hi = srl(n, I32(16))
        n = n_hi + (n & 0xFFFF)
        size, bad = size + n, bad | n
        lo = srl(lo, n) | sll(hi, n ^ 31)
        hi = srl(hi, n) | top | srl(top, n_hi)
    far = size >= 32
    string = [jnp.where(far, u, w) for u, w in zip([0] + string, string)]
    string = _shift_right(string, size & 31)
    string[0], string[1] = string[0] | hi, string[1] | sll(lo, I32(1))
    bad = bad | srl(size + 1, I32(1))
    return codes, (string, total + size, bad)


def _encode_finish(window, state, tmp):
    base, rank, above = window
    string, total, bad = state
    total = total + above
    bad = (srl(bad | above, I32(5)) != 0) | (total > 32 * RUN)
    string = _shift_right(string, (above - 1) & 31)
    end = _running_sum(total + _header_bits())
    start = end - total
    string = _shift_right(string + [_splat(0)], start & 31) + [_splat(0)] * (7 - RUN)
    for j, w in enumerate(string):
        tmp[:, pl.ds(8 * j, 8)] = w
    first = srl(start, I32(5))
    pool = [_splat(0)] * len(POOL)
    for s in range(8):
        q = _row(first, s)
        w = _rotate(tmp[:, pl.ds(s, 8, stride=8)], q, up=False)
        at = srl(q + ((_sublane() - q) & 7), I32(3))
        pool = [v | jnp.where(at == j, w, 0) for j, v in enumerate(pool)]
    need = jnp.where(bad, 2000, end).astype(jnp.float32)
    need = [jnp.max(need[h]) for h in range(2)]
    level = [(v > 3 * 256).astype(I32) + (v > 4 * 256).astype(I32) for v in need]
    header = sll(base, I32(22)) | sll(rank, I32(19))
    pool[0] = pool[0] | jnp.where(_header_bits() != 0, header, 0)
    return pool, level


def _decode_start(codes, pool, header, tmp):
    ones = _splat(1)
    for v in codes:
        ones = ones + lax.population_count(~(v | srl(v, I32(1))) & _i(0x55555555))
    before = _running_sum(ones) - ones
    pool = [srl(sll(pool[0], _header_bits()), _header_bits())] + pool[1:]
    first = passed = upto = _splat(0)
    for v in pool:
        seen = _running_sum(lax.population_count(v)) + upto
        for s in range(8):
            upto = _row(seen, s)
            ok = upto < before
            first, passed = jnp.where(ok, first + 1, first), jnp.where(ok, upto, passed)
    for s in range(8):
        q = _row(first, s)
        at = srl(q + ((_sublane() - q) & 7), I32(3))
        w = _splat(0)
        for j, v in enumerate(pool):
            w = jnp.where(at == j, v, w)
        tmp[:, pl.ds(8 * s, 8)] = _rotate(w, q, up=True)
    string = [tmp[:, pl.ds(j, 8, stride=8)] for j in range(RUN + 2)]
    left, w, skip = before - passed, string[0], _splat(0)
    for d in (16, 8, 4, 2, 1):
        c = lax.population_count(srl(w, I32(32 - d)))
        ok = c < left
        left, skip = jnp.where(ok, left - c, left), jnp.where(ok, skip + d, skip)
        w = jnp.where(ok, sll(w, I32(d)), w)
    opening = _sublane() == 0
    string = _shift_left(string, jnp.where(opening, _header_bits(), skip))[: RUN + 1]
    lead = lax.clz(jnp.where(opening, string[0], string[0] & _i(0x7FFFFFFF)) | 1)
    above = jnp.where(opening, lead + 1, lead)
    base, rank = srl(header, I32(22)) & 255, srl(header, I32(19)) & 7
    return (base, rank, above), _shift_left(string, lead)[:RUN]


def _decode_group(codes, window, string):
    base, rank, above = window
    roof = sll(_both(base + 4), I32(7))
    hi, lo = string[0], sll(string[0], I32(31)) | srl(string[1], I32(1))
    size, es = _splat(0), []
    for i in range(8):
        e, took = roof, []
        for at, to in ((16 + 2 * i, 23), (2 * i, 7)):
            code = srl(codes, I32(at)) & 3
            n = lax.clz(hi & _i(0x7FFFFFFF))
            u = rank - n
            drop = jnp.where(u > -above, jnp.where(u > 0, n + 3, u), n + (3 - above))
            e = e - sll(jnp.where(code == 0, drop, code), I32(to))
            took.append(jnp.where(code == 0, n, 0))
            hi = sll(hi, took[-1])
        n = took[0] + took[1]
        hi, lo = hi | srl(lo, n ^ 31), sll(lo, n)
        size = size + n
        es.append(e)
    far = size >= 32
    string = [jnp.where(far, u, w) for w, u in zip(string, string[1:] + [0])]
    es = [jnp.concatenate(es[i : i + 4], axis=2) for i in (0, 4)]
    return jnp.concatenate(es, axis=1), _shift_left(string, size & 31)


def _rows(r, n, unit=16):
    return pl.ds(r if isinstance(r, int) else pl.multiple_of(r, unit), n)


def _pairs(r, n):
    return _rows(r // 2, n // 2, 8)


def _plain_slot(j):
    return j + 1 + (j + 1 >= POOL[0]).astype(I32)


def pallas_dist_ar_i_i_m2048_n512_kernel(x: jax.Array):
    cuts = [[(sum(c[:k]), n) for k, n in enumerate(c)] for c in CUTS]
    sem0 = [sum(len(c) + len(LEVELS) for c in CUTS[:b]) for b in range(7)]

    def body(x_hbm, out, x_give, x_keep, x_far, via, exps, peaks, decoded, tmp,
             bytes_out, bytes_in, exps_out, exps_in, levels, ld, snd, rcv, ready):
        p = lax.axis_index("i")
        odd = p & 1
        half = [(p == 3).astype(I32) ^ h for h in range(2)]
        nbr = [p ^ (1 + 2 * v) for v in half]
        bit = [jnp.where(v == 0, (p ^ (p >> 1)) & 1, p >> 1) for v in half]
        keep = [(2 * half[h] + bit[h]) * Q for h in range(2)]
        give = [(2 * half[h] + 1 - bit[h]) * Q for h in range(2)]

        def signal(sem):
            for to in nbr[::-1]:
                pl.semaphore_signal(sem, 1, device_id=(to,), device_id_type=pl.DeviceIdType.MESH)

        def load(dst, base, k, r, n):
            return [
                pltpu.make_async_copy(
                    x_hbm.at[_rows(base[h] + r, n)], dst.at[h, pl.ds(r, n)], ld.at[2 * k + h])
                for h in range(2)
            ]

        def remote(src, dst, k, h, to, incoming):
            there = h if incoming else half[h] ^ (to == 3).astype(I32)
            return pltpu.make_async_remote_copy(
                src, dst(there), snd.at[2 * k + h], rcv.at[2 * k + there],
                device_id=(to,), device_id_type=pl.DeviceIdType.MESH)

        def block_copy(src, dst, b, h, part, k, incoming):
            return remote(src.at[b, h, part], lambda j: dst.at[b, j, part], sem0[b] + k,
                          h, nbr[h ^ (b // 2 == 1)], incoming)

        def with_copy(copy, act, h, incoming, has_rerouted_rows):
            if has_rerouted_rows:
                short = p == 0 if incoming else odd > h
                pl.when(short)(lambda: act(copy(1)))
                pl.when(~short)(lambda: act(copy(0)))
            else:
                act(copy(0))

        def with_exp_copy(b, h, level, act, incoming=False):
            def copy(omit):
                part = pl.ds(LEVELS[level][0] + omit, LEVELS[level][1] - omit)
                return block_copy(exps_out, exps_in, b, h, part, level, incoming)

            with_copy(copy, act, h, incoming, (b, level) == (1, 0))

        def with_byte_copy(b, h, k, act, incoming=False):
            def copy(omit):
                part = _pairs(cuts[b][k][0], cuts[b][k][1] - omit * ROUND)
                return block_copy(bytes_out, bytes_in, b, h, part, len(LEVELS) + k, incoming)

            with_copy(copy, act, h, incoming, (b, k) == (1, len(cuts[1]) - 1))

        def with_exp_copies(b, h, first, level, act, incoming=False):
            if first == 0:
                with_exp_copy(b, h, 0, act, incoming)
            for k in range(1, len(LEVELS)):
                pl.when(level >= k)(lambda: with_exp_copy(b, h, k, act, incoming))

        start = lambda d: d.start()
        sent = lambda d: d.wait_send()
        landed = lambda d: d.wait_recv()

        def detour(h, incoming=False):
            return remote(via.at[2], lambda j: via.at[j], sem0[6], h, nbr[1], incoming)

        def send_bytes(b, h, k):
            with_byte_copy(b, h, k, start)

        def wait_bytes(b, ks):
            for k in ks:
                for h in range(2):
                    with_byte_copy(b, h, k, landed, incoming=True)

        def stage(b, hs, r, v):
            n = v.shape[1]
            e, m = _split(v)
            bytes_out[b, hs, _pairs(r, n)] = m
            exps[hs, _pairs(r, n)] = srl(e, I32(7))
            hi, lo = (lax.bitcast_convert_type(u, jnp.float32)
                      for u in (srl(e, I32(1)), sll(e, I32(15))))
            t = jnp.maximum(hi, lo)
            t = jnp.maximum(t[..., :256], t[..., 256:])
            peaks[hs, _pairs(r, n)] = jnp.maximum(t[..., :128], t[..., 128:])

        def each_64_rows(f, then_send=None):
            @pl.loop(0, B // 64, unroll=True)
            def _(t):
                f(t * 64)
                for k in range(FRONT[then_send] if then_send else 0):
                    @pl.when(t == sum(cuts[then_send][k]) // 64 - 1)
                    def _():
                        for h in range(2):
                            send_bytes(then_send, h, k)

        def encode_and_send(b, base, rank):
            t, n = peaks[...], B // 2
            while n > 8:
                n //= 2
                t = jnp.maximum(t[:, :n], t[:, n:])
            top = srl(lax.bitcast_convert_type(t, I32), I32(22))
            window = (base, rank, jnp.where(top > base + 4, top - base - 3, 1))
            if b == 1:
                @pl.when(odd == 1)
                def _():
                    filler = _both(base[0] + 1)
                    exps[0, _pairs(B - ROUND, ROUND)] = jnp.tile(filler, (ROUND // 16, N // 128))

            def group(j, state):
                exps_out[b, :, j], state = _encode_group(
                    exps[:, _pairs(32 * (GROUPS - 1 - j), 32)], window, state)
                return state

            state = ([_splat(0)] * RUN, _splat(0), _splat(0))
            state = lax.fori_loop(0, GROUPS, group, state, unroll=True)
            pool, level = _encode_finish(window, state, tmp)
            for at, v in zip(POOL[1:], pool[1:]):
                exps_out[b, :, at] = v
            for h in range(2):
                corner = jnp.where(_header_bits()[h] != 0, sll(level[h], I32(30)), 0)
                exps_out[b, h, POOL[0]] = pool[0][h] | corner
                levels[2 * b + h] = level[h]

                @pl.when(level[h] == 2)
                def _():
                    exps_out[b, h, POOL[0]] = corner

                    @pl.loop(0, B // 16)
                    def _(j):
                        e = exps[h, _pairs(16 * j, 16)]
                        e = e[:, :256] | sll(e[:, 256:], I32(8))
                        exps_out[b, h, _plain_slot(2 * j)] = e[:, :128]
                        exps_out[b, h, _plain_slot(2 * j + 1)] = e[:, 128:]

                with_exp_copies(b, h, 0, level[h], start)
                for k in range(FRONT[b], len(cuts[b])):
                    send_bytes(b, h, k)

        def wait_and_decode(b):
            for h in range(2):
                with_exp_copy(b, h, 0, landed, incoming=True)
            if b == 1:
                @pl.when(p == 0)
                def _():
                    exps_in[1, :, 0] = _splat(0xFFFFFFFF)

            header = [exps_in[b, h, POOL[0], 0, 0] for h in range(2)]
            level = [srl(v, I32(30)) for v in header]
            for h in range(2):
                @pl.when(level[h] == 0)
                def _():
                    exps_in[b, h, POOL[-1]] = jnp.zeros((8, 128), I32)

                with_exp_copies(b, h, 1, level[h], landed, incoming=True)

            @pl.when((level[0] < 2) | (level[1] < 2))
            def _():
                use = [jnp.where(level[h] < 2, h, 1 - h) for h in range(2)]
                head = [jnp.where(level[h] < 2, header[h], header[1 - h]) for h in range(2)]
                vreg = lambda at: jnp.stack([exps_in[b, use[h], at] for h in range(2)])
                window, string = _decode_start(
                    [vreg(j) for j in range(GROUPS)], [vreg(at) for at in POOL],
                    jnp.stack([jnp.full((8, 128), v, I32) for v in head]), tmp)

                def group(g, string):
                    decoded[:, _pairs(32 * g, 32)], string = _decode_group(
                        vreg(GROUPS - 1 - g), window, string)
                    return string

                lax.fori_loop(0, GROUPS, group, string, unroll=True)

            for h in range(2):
                @pl.when(level[h] == 2)
                def _():
                    @pl.loop(0, B // 16)
                    def _(j):
                        v = [exps_in[b, h, _plain_slot(2 * j + k)] for k in range(2)]
                        v = [sll(u, I32(7)) for u in v] + [srl(u, I32(1)) for u in v]
                        decoded[h, _pairs(16 * j, 16)] = jnp.concatenate(v, axis=1) & _i(0x7F807F80)

        def received(b, r, n):
            return _join(decoded[:, _pairs(r, n)], bytes_in[b, :, _pairs(r, n)])

        def write(base, r, v):
            for h in range(2):
                out[_rows(base[h] + r, v.shape[1])] = v[h]

        def wait_sent(b):
            for h in range(2):
                for k in range(len(cuts[b])):
                    with_byte_copy(b, h, k, sent)
                with_exp_copies(b, h, 0, levels[2 * b + h], sent)

        give_loads = [load(x_give, give, k, r, n) for k, (r, n) in enumerate(cuts[0] + [(B, B)])]
        keep_loads = [load(x_keep, keep, len(give_loads) + k, k * B, B) for k in range(2)]
        far_load = pltpu.make_async_copy(
            x_hbm.at[_rows(give[0] + Q - ROUND, ROUND)], x_far, ld.at[2 * len(give_loads) + 4])

        barrier = pltpu.get_barrier_semaphore()
        pl.when(p != 2)(lambda: signal(barrier))
        give_loads[0][0].start()

        @pl.when(p == 2)
        def _():
            pl.semaphore_wait(barrier, 2)
            signal(ready)

        early = sum(give_loads[:-1], [])
        early.insert(2 * LATE + 2, far_load)
        for d in early[1:]:
            d.start()
        pl.when(p == 0)(lambda: pl.semaphore_wait(barrier, 2))
        pl.when(odd == 1)(lambda: pl.semaphore_wait(barrier, 1))

        for k, (r, n) in enumerate(cuts[0]):
            for h in range(2):
                give_loads[k][h].wait()
                stage(0, pl.ds(h, 1), r, x_give[pl.ds(h, 1), pl.ds(r, n)])
                if h == 0 or k >= LATE:
                    send_bytes(0, h, k)
                else:
                    pl.when(odd == 0)(lambda: send_bytes(0, 1, k))
                if k == 0:
                    give_loads[-1][h].start()
                if (k, h) == (LATE, 0):
                    base, rank = _pick_window(exps[:, :8])

                    @pl.when(odd == 1)
                    def _():
                        pl.semaphore_wait(ready, 1)
                        for j in range(LATE):
                            send_bytes(0, 1, j)

                if (k, h) == (LATE, 1):
                    far_load.wait()

                    @pl.when(odd == 1)
                    def _():
                        via[2] = x_far[...].astype(jnp.bfloat16)
                        detour(0).start()

        for d in keep_loads[0]:
            d.start()
        encode_and_send(0, base, rank)
        for d in keep_loads[1]:
            d.start()
        for d in give_loads[-1]:
            d.wait()
        both = slice(None)
        each_64_rows(lambda r: stage(1, both, r, x_give[:, _rows(B + r, 64)]), then_send=1)

        @pl.when(p == 2)
        def _():
            for h in range(2):
                detour(h, incoming=True).wait_recv()
            t = x_give[:, pl.ds(Q - ROUND, ROUND)] + via[:2].astype(jnp.float32)
            stage(1, both, B - ROUND, t)

        encode_and_send(1, *_pick_window(exps[:, :8]))

        for b in range(4):
            r0 = b % 2 * B
            wait_and_decode(b)
            wait_bytes(b, range(len(cuts[b])))
            if b < 2:
                for d in keep_loads[b]:
                    d.wait()
            if b == 1:
                @pl.when(p == 0)
                def _():
                    gone = _pairs(B - ROUND, ROUND)
                    bytes_in[1, :, gone] = jnp.zeros((2, ROUND // 2, N // 2), I32)
                    decoded[:, gone] = jnp.zeros((2, ROUND // 2, N), I32)

            def add(r):
                t = x_keep[:, _rows(r0 + r, 64)] + received(b, r, 64).astype(jnp.float32)
                if b < 2:
                    x_keep[:, _rows(r0 + r, 64)] = t
                else:
                    write(keep, r0 + r, t.astype(jnp.bfloat16))
                stage(b + 2, both, r, t)

            each_64_rows(add, then_send=b + 2)
            encode_and_send(b + 2, *_pick_window(exps[:, :8]))

        wait_and_decode(4)
        wait_bytes(4, range(len(cuts[4])))
        each_64_rows(lambda r: write(give, r, received(4, r, 64)))
        for b in range(5):
            wait_sent(b)
        pl.when(odd == 1)(lambda: detour(0).wait_send())
        wait_and_decode(5)
        for k, (r, n) in enumerate(cuts[5]):
            if k == len(cuts[5]) - 1:
                wait_sent(5)
            wait_bytes(5, [k])
            write(give, B + r, received(5, r, n))

    f32, vmem, dma = jnp.float32, pltpu.VMEM, pltpu.SemaphoreType.DMA
    return pl.pallas_call(
        body,
        out_shape=vmem((M, N), jnp.bfloat16),
        in_specs=[pl.BlockSpec(memory_space=pltpu.HBM)],
        out_specs=pl.BlockSpec(memory_space=vmem),
        scratch_shapes=[
            vmem((2, Q, N), f32),
            vmem((2, Q, N), f32),
            vmem((ROUND, N), f32),
            vmem((3, ROUND, N), jnp.bfloat16),
            vmem((2, B // 2, N), I32),
            vmem((2, B // 2, 128), f32),
            vmem((2, B // 2, N), I32),
            vmem((2, 72, 128), I32),
            vmem((6, 2, B // 2, N // 2), I32),
            vmem((6, 2, B // 2, N // 2), I32),
            vmem((6, 2, sum(LEVELS[-1]), 8, 128), I32),
            vmem((6, 2, sum(LEVELS[-1]), 8, 128), I32),
            pltpu.SMEM((12,), I32),
            dma((2 * len(CUTS[0]) + 8,)),
            dma((2 * sem0[6] + 2,)),
            dma((2 * sem0[6] + 2,)),
            pltpu.SemaphoreType.REGULAR,
        ],
        compiler_params=pltpu.CompilerParams(collective_id=0, disable_semaphore_checks=True),
    )(x)
```

```python
import jax
import jax.numpy as jnp
from jax import lax
from jax.experimental import pallas as pl
from jax.experimental.pallas import tpu as pltpu

M, N = 2048, 512
Q = M // 4
B = Q // 2
GROUPS = B // 32

CUTS = (
    (16, 16, 32, 48, 64, 48, 32),
    (128, 128),
    (64, 128, 64),
    (128, 128),
    (128, 128),
    (64, 96, 64, 16, 16),
)
FRONT = (7, 1, 2, 1, 1, 1)
LATE = 3
ROUND = 32

POOL = (8, 9, 10, 11)
LEVELS = ((0, 11), (11, 1), (12, 22))
RUN = 6
HEADER = 13

I32 = jnp.int32
srl, sll = lax.shift_right_logical, lax.shift_left
VREGS = (2, 8, 128)


def _i(v):
    return I32(v - (1 << 32) if v >= (1 << 31) else v)


def _splat(v):
    return jnp.full(VREGS, _i(v), I32)


def _sublane():
    return lax.broadcasted_iota(I32, VREGS, 1)


def _header_bits():
    lane = lax.broadcasted_iota(I32, VREGS, 2)
    return jnp.where((_sublane() == 0) & (lane == 0), HEADER, 0)


def _level_bits(level):
    return jnp.where(_header_bits()[0] != 0, sll(level, I32(30)), 0)


def _row(v, s):
    return jnp.broadcast_to(v[:, s : s + 1], VREGS)


def _both(v):
    return sll(v, I32(16)) | v


def _running_sum(v):
    for d in (1, 2, 4):
        v = v + jnp.where(_sublane() >= d, pltpu.roll(v, d, 1), 0)
    return v


def _rotate(v, n, up):
    for d in (1, 2, 4):
        v = jnp.where((n & d) != 0, pltpu.roll(v, 8 - d if up else d, 1), v)
    return v


def _shift_right(ws, n):
    rest = [srl(w, n) | sll(sll(u, I32(1)), n ^ 31) for u, w in zip(ws, ws[1:])]
    return [srl(ws[0], n)] + rest


def _shift_left(ws, n):
    rest = [sll(w, n) | srl(srl(u, I32(1)), n ^ 31) for w, u in zip(ws, ws[1:])]
    return rest + [sll(ws[-1], n)]


def _split(v):
    w = pltpu.bitcast(v.astype(jnp.bfloat16), I32)
    a, b = w[..., : N // 2], w[..., N // 2 :]
    rest = sll(b & _i(0x007F007F), I32(7)) | srl(b & _i(0x80008000), I32(1))
    return w & _i(0x7F807F80), (a & _i(0x807F807F)) | rest


def _join(e, m):
    b = (srl(m, I32(7)) & _i(0x007F007F)) | (sll(m, I32(1)) & _i(0x80008000))
    w = jnp.concatenate([m & _i(0x807F807F), b], axis=-1) | e
    return pltpu.bitcast(w, jnp.bfloat16)


def _pick_window(sample):
    t = sum(sample[..., j : j + 128] for j in range(0, N, 128))
    t = (srl(t, I32(16)) + (t & 0xFFFF)).astype(jnp.float32)
    t = jnp.sum(jnp.sum(t, axis=2, keepdims=True), axis=1, keepdims=True)
    mean = jnp.broadcast_to(t, VREGS) * (1.0 / (16 * N)) + 0.12
    whole = mean.astype(I32)
    rank = (7.9 - 6.3 * (mean - whole.astype(jnp.float32))).astype(I32)
    return jnp.clip(whole - 1, 0, 251), jnp.clip(rank, 1, 7)


def _peak(e):
    hi, lo = (lax.bitcast_convert_type(u, jnp.float32)
              for u in (srl(e, I32(1)), sll(e, I32(15))))
    t = jnp.maximum(hi, lo)
    t = jnp.maximum(t[..., :256], t[..., 256:])
    return jnp.maximum(t[..., :128], t[..., 128:])


def _encode_start(base, rank, peak):
    while peak.shape[1] > 8:
        n = peak.shape[1] // 2
        peak = jnp.maximum(peak[:, :n], peak[:, n:])
    top = srl(lax.bitcast_convert_type(peak, I32), I32(22))
    window = (base, rank, jnp.where(top > base + 4, top - base - 3, 1))
    return window, ([_splat(0)] * RUN, _splat(0), _splat(0))


def _plain(e):
    e = e[:, :256] | sll(e[:, 256:], I32(8))
    return e[:, :128], e[:, 128:]


def _unplain(vs):
    vs = [sll(v, I32(7)) for v in vs] + [srl(v, I32(1)) for v in vs]
    return jnp.concatenate(vs, axis=1) & _i(0x7F807F80)


def _encode_group(es, window, state):
    base, rank, above = window
    string, total, bad = state
    guard, top = _i(0x80008000), _splat(1 << 31)
    fence_lo, fence_hi = _both(base) | guard, guard - _both(base + 4)
    rank2, skip2, above2 = _both(rank), _both(rank - 1), _both(above)
    hi, lo = top, _splat(0)
    size = codes = _splat(0)
    for i in reversed(range(8)):
        e = es[:, i // 4 * 8 : i // 4 * 8 + 8, i % 4 * 128 : i % 4 * 128 + 128]
        t = fence_lo - e
        g = t & guard
        one = srl(g, I32(15))
        low = g - one
        g = (t - skip2) & guard
        skip = above2 & (g - srl(g, I32(15)))
        u = e + fence_hi
        g = u & guard
        high = g - srl(g, I32(15))
        n = (t & low) + one + skip + ((u + rank2) & high)
        codes = codes | sll(t & _i(0x00030003) & ~(low | high), I32(2 * i))
        n_hi = srl(n, I32(16))
        n = n_hi + (n & 0xFFFF)
        size, bad = size + n, bad | n
        lo = srl(lo, n) | sll(hi, n ^ 31)
        hi = srl(hi, n) | top | srl(top, n_hi)
    far = size >= 32
    string = [jnp.where(far, u, w) for u, w in zip([0] + string, string)]
    string = _shift_right(string, size & 31)
    string[0], string[1] = string[0] | hi, string[1] | sll(lo, I32(1))
    bad = bad | srl(size + 1, I32(1))
    return codes, (string, total + size, bad)


def _encode_finish(window, state, tmp, sizes):
    base, rank, above = window
    string, total, bad = state
    total = total + above
    bad = (srl(bad | above, I32(5)) != 0) | (total > 32 * RUN)
    string = _shift_right(string, (above - 1) & 31)
    end = _running_sum(total + _header_bits())
    start = end - total
    string = _shift_right(string + [_splat(0)], start & 31) + [_splat(0)] * (7 - RUN)
    for j, w in enumerate(string):
        tmp[:, pl.ds(8 * j, 8)] = w
    first = srl(start, I32(5))
    pool = [_splat(0)] * sizes[1]
    for s in range(8):
        q = _row(first, s)
        w = _rotate(tmp[:, pl.ds(s, 8, stride=8)], q, up=False)
        at = srl(q + ((_sublane() - q) & 7), I32(3))
        pool = [v | jnp.where(at == j, w, 0) for j, v in enumerate(pool)]
    need = jnp.where(bad, 2000, end).astype(jnp.float32)
    need = [jnp.max(need[h]) for h in range(2)]
    level = [sum((v > 256 * n).astype(I32) for n in sizes) for v in need]
    header = sll(base, I32(22)) | sll(rank, I32(19))
    pool[0] = pool[0] | jnp.where(_header_bits() != 0, header, 0)
    return pool, level


def _decode_start(codes, pool, header, tmp):
    ones = _splat(1)
    for v in codes:
        ones = ones + lax.population_count(~(v | srl(v, I32(1))) & _i(0x55555555))
    before = _running_sum(ones) - ones
    pool = [srl(sll(pool[0], _header_bits()), _header_bits())] + pool[1:]
    first = passed = upto = _splat(0)
    for v in pool:
        seen = _running_sum(lax.population_count(v)) + upto
        for s in range(8):
            upto = _row(seen, s)
            ok = upto < before
            first, passed = jnp.where(ok, first + 1, first), jnp.where(ok, upto, passed)
    for s in range(8):
        q = _row(first, s)
        at = srl(q + ((_sublane() - q) & 7), I32(3))
        w = _splat(0)
        for j, v in enumerate(pool):
            w = jnp.where(at == j, v, w)
        tmp[:, pl.ds(8 * s, 8)] = _rotate(w, q, up=True)
    string = [tmp[:, pl.ds(j, 8, stride=8)] for j in range(RUN + 2)]
    left, w, skip = before - passed, string[0], _splat(0)
    for d in (16, 8, 4, 2, 1):
        c = lax.population_count(srl(w, I32(32 - d)))
        ok = c < left
        left, skip = jnp.where(ok, left - c, left), jnp.where(ok, skip + d, skip)
        w = jnp.where(ok, sll(w, I32(d)), w)
    opening = _sublane() == 0
    string = _shift_left(string, jnp.where(opening, _header_bits(), skip))[: RUN + 1]
    lead = lax.clz(jnp.where(opening, string[0], string[0] & _i(0x7FFFFFFF)) | 1)
    above = jnp.where(opening, lead + 1, lead)
    base, rank = srl(header, I32(22)) & 255, srl(header, I32(19)) & 7
    return (base, rank, above), _shift_left(string, lead)[:RUN]


def _decode_group(codes, window, string):
    base, rank, above = window
    roof = sll(_both(base + 4), I32(7))
    hi, lo = string[0], sll(string[0], I32(31)) | srl(string[1], I32(1))
    size, es = _splat(0), []
    for i in range(8):
        e, took = roof, []
        for at, to in ((16 + 2 * i, 23), (2 * i, 7)):
            code = srl(codes, I32(at)) & 3
            n = lax.clz(hi & _i(0x7FFFFFFF))
            u = rank - n
            drop = jnp.where(u > -above, jnp.where(u > 0, n + 3, u), n + (3 - above))
            e = e - sll(jnp.where(code == 0, drop, code), I32(to))
            took.append(jnp.where(code == 0, n, 0))
            hi = sll(hi, took[-1])
        n = took[0] + took[1]
        hi, lo = hi | srl(lo, n ^ 31), sll(lo, n)
        size = size + n
        es.append(e)
    far = size >= 32
    string = [jnp.where(far, u, w) for w, u in zip(string, string[1:] + [0])]
    es = [jnp.concatenate(es[i : i + 4], axis=2) for i in (0, 4)]
    return jnp.concatenate(es, axis=1), _shift_left(string, size & 31)


def _rows(r, n, unit=16):
    return pl.ds(r if isinstance(r, int) else pl.multiple_of(r, unit), n)


def _pairs(r, n):
    return _rows(r // 2, n // 2, 8)


def _plain_slot(j):
    return j + 1 + (j + 1 >= POOL[0]).astype(I32)


def pallas_dist_ar_i_i_m2048_n512_kernel(x: jax.Array):
    cuts = [[(sum(c[:k]), n) for k, n in enumerate(c)] for c in CUTS]
    sem0 = [sum(len(c) + len(LEVELS) for c in CUTS[:b]) for b in range(7)]

    def body(x_hbm, out, x_give, x_keep, x_far, via_bytes, via_exps, exps, peaks, decoded, tmp,
             bytes_out, bytes_in, exps_out, exps_in, levels, ld, snd, rcv, ready):
        p = lax.axis_index("i")
        odd = p & 1
        half = [(p == 3).astype(I32) ^ h for h in range(2)]
        nbr = [p ^ (1 + 2 * v) for v in half]
        bit = [jnp.where(v == 0, (p ^ (p >> 1)) & 1, p >> 1) for v in half]
        keep = [(2 * half[h] + bit[h]) * Q for h in range(2)]
        give = [(2 * half[h] + 1 - bit[h]) * Q for h in range(2)]

        def signal(sem):
            for to in nbr[::-1]:
                pl.semaphore_signal(sem, 1, device_id=(to,), device_id_type=pl.DeviceIdType.MESH)

        def load(dst, base, k, r, n):
            return [
                pltpu.make_async_copy(
                    x_hbm.at[_rows(base[h] + r, n)], dst.at[h, pl.ds(r, n)], ld.at[2 * k + h])
                for h in range(2)
            ]

        def remote(src, dst, k, h, to, incoming):
            there = h if incoming else half[h] ^ (to == 3).astype(I32)
            return pltpu.make_async_remote_copy(
                src, dst(there), snd.at[2 * k + h], rcv.at[2 * k + there],
                device_id=(to,), device_id_type=pl.DeviceIdType.MESH)

        def block_copy(src, dst, b, h, part, k, incoming):
            return remote(src.at[b, h, part], lambda j: dst.at[b, j, part], sem0[b] + k,
                          h, nbr[h ^ (b // 2 == 1)], incoming)

        def with_copy(copy, act, h, incoming, has_rerouted_rows):
            if has_rerouted_rows:
                short = p == 0 if incoming else odd > h
                pl.when(short)(lambda: act(copy(1)))
                pl.when(~short)(lambda: act(copy(0)))
            else:
                act(copy(0))

        def with_exp_copy(b, h, level, act, incoming=False):
            def copy(omit):
                part = pl.ds(LEVELS[level][0] + omit, LEVELS[level][1] - omit)
                return block_copy(exps_out, exps_in, b, h, part, level, incoming)

            with_copy(copy, act, h, incoming, (b, level) == (1, 0))

        def with_byte_copy(b, h, k, act, incoming=False):
            def copy(omit):
                part = _pairs(cuts[b][k][0], cuts[b][k][1] - omit * ROUND)
                return block_copy(bytes_out, bytes_in, b, h, part, len(LEVELS) + k, incoming)

            with_copy(copy, act, h, incoming, (b, k) == (1, len(cuts[1]) - 1))

        def with_exp_copies(b, h, first, level, act, incoming=False):
            if first == 0:
                with_exp_copy(b, h, 0, act, incoming)
            for k in range(1, len(LEVELS)):
                pl.when(level >= k)(lambda: with_exp_copy(b, h, k, act, incoming))

        start = lambda d: d.start()
        sent = lambda d: d.wait_send()
        landed = lambda d: d.wait_recv()

        def detour(h, k, incoming=False):
            ref, part = ((via_bytes, slice(None)), (via_exps, pl.ds(0, 2)), (via_exps, pl.ds(2, 4)))[k]
            return remote(ref.at[2, part], lambda j: ref.at[j, part], sem0[6] + k, h, nbr[1], incoming)

        def send_bytes(b, h, k):
            with_byte_copy(b, h, k, start)

        def wait_bytes(b, ks):
            for k in ks:
                for h in range(2):
                    with_byte_copy(b, h, k, landed, incoming=True)

        def stage(b, hs, r, v):
            n = v.shape[1]
            e, m = _split(v)
            bytes_out[b, hs, _pairs(r, n)] = m
            exps[hs, _pairs(r, n)] = srl(e, I32(7))
            peaks[hs, _pairs(r, n)] = _peak(e)

        def each_64_rows(f, then_send=None):
            @pl.loop(0, B // 64, unroll=True)
            def _(t):
                f(t * 64)
                for k in range(FRONT[then_send] if then_send else 0):
                    @pl.when(t == sum(cuts[then_send][k]) // 64 - 1)
                    def _():
                        for h in range(2):
                            send_bytes(then_send, h, k)

        def encode_and_send(b, base, rank):
            window, state = _encode_start(base, rank, peaks[...])
            if b == 1:
                @pl.when(odd == 1)
                def _():
                    filler = _both(base[0] + 1)
                    exps[0, _pairs(B - ROUND, ROUND)] = jnp.tile(filler, (ROUND // 16, N // 128))

            def group(j, state):
                exps_out[b, :, j], state = _encode_group(
                    exps[:, _pairs(32 * (GROUPS - 1 - j), 32)], window, state)
                return state

            state = lax.fori_loop(0, GROUPS, group, state, unroll=True)
            pool, level = _encode_finish(window, state, tmp, (3, 4))
            for at, v in zip(POOL[1:], pool[1:]):
                exps_out[b, :, at] = v
            for h in range(2):
                corner = _level_bits(level[h])
                exps_out[b, h, POOL[0]] = pool[0][h] | corner
                levels[2 * b + h] = level[h]

                @pl.when(level[h] == 2)
                def _():
                    exps_out[b, h, POOL[0]] = corner

                    @pl.loop(0, B // 16)
                    def _(j):
                        for k, v in enumerate(_plain(exps[h, _pairs(16 * j, 16)])):
                            exps_out[b, h, _plain_slot(2 * j + k)] = v

                with_exp_copies(b, h, 0, level[h], start)
                for k in range(FRONT[b], len(cuts[b])):
                    send_bytes(b, h, k)

        def decode(msg, header, groups, pool):
            coded = [srl(v, I32(30)) < 2 for v in header]

            @pl.when(coded[0] | coded[1])
            def _():
                use = [jnp.where(coded[h], h, 1 - h) for h in range(2)]
                head = [jnp.where(coded[h], header[h], header[1 - h]) for h in range(2)]
                vreg = lambda at: jnp.stack([msg[use[h], at] for h in range(2)])
                window, string = _decode_start(
                    [vreg(j) for j in range(groups)], [vreg(at) for at in pool],
                    jnp.stack([jnp.full((8, 128), v, I32) for v in head]), tmp)

                def group(g, string):
                    decoded[:, _pairs(32 * g, 32)], string = _decode_group(
                        vreg(groups - 1 - g), window, string)
                    return string

                lax.fori_loop(0, groups, group, string, unroll=True)

        def wait_and_decode(b):
            for h in range(2):
                with_exp_copy(b, h, 0, landed, incoming=True)
            if b == 1:
                @pl.when(p == 0)
                def _():
                    exps_in[1, :, 0] = _splat(0xFFFFFFFF)

            header = [exps_in[b, h, POOL[0], 0, 0] for h in range(2)]
            level = [srl(v, I32(30)) for v in header]
            for h in range(2):
                @pl.when(level[h] == 0)
                def _():
                    exps_in[b, h, POOL[-1]] = jnp.zeros((8, 128), I32)

                with_exp_copies(b, h, 1, level[h], landed, incoming=True)

            decode(exps_in.at[b], header, GROUPS, POOL)
            for h in range(2):
                @pl.when(level[h] == 2)
                def _():
                    @pl.loop(0, B // 16)
                    def _(j):
                        decoded[h, _pairs(16 * j, 16)] = _unplain(
                            [exps_in[b, h, _plain_slot(2 * j + k)] for k in range(2)])

        def received(b, r, n):
            return _join(decoded[:, _pairs(r, n)], bytes_in[b, :, _pairs(r, n)])

        def write(base, r, v):
            for h in range(2):
                out[_rows(base[h] + r, v.shape[1])] = v[h]

        def wait_sent(b):
            for h in range(2):
                for k in range(len(cuts[b])):
                    with_byte_copy(b, h, k, sent)
                with_exp_copies(b, h, 0, levels[2 * b + h], sent)

        give_loads = [load(x_give, give, k, r, n) for k, (r, n) in enumerate(cuts[0] + [(B, B)])]
        keep_loads = [load(x_keep, keep, len(give_loads) + k, k * B, B) for k in range(2)]
        far_load = pltpu.make_async_copy(
            x_hbm.at[_rows(give[0] + Q - ROUND, ROUND)], x_far, ld.at[2 * len(give_loads) + 4])

        barrier = pltpu.get_barrier_semaphore()
        pl.when(p != 2)(lambda: signal(barrier))
        give_loads[0][0].start()

        @pl.when(p == 2)
        def _():
            pl.semaphore_wait(barrier, 2)
            signal(ready)

        early = sum(give_loads[:-1], [])
        early.insert(2 * LATE + 2, far_load)
        for d in early[1:]:
            d.start()
        pl.when(p == 0)(lambda: pl.semaphore_wait(barrier, 2))
        pl.when(odd == 1)(lambda: pl.semaphore_wait(barrier, 1))

        for k, (r, n) in enumerate(cuts[0]):
            for h in range(2):
                give_loads[k][h].wait()
                stage(0, pl.ds(h, 1), r, x_give[pl.ds(h, 1), pl.ds(r, n)])
                if h == 0 or k >= LATE:
                    send_bytes(0, h, k)
                else:
                    pl.when(odd == 0)(lambda: send_bytes(0, 1, k))
                if k == 0:
                    give_loads[-1][h].start()
                if (k, h) == (LATE, 0):
                    base, rank = _pick_window(exps[:, :8])

                    @pl.when(odd == 1)
                    def _():
                        pl.semaphore_wait(ready, 1)
                        for j in range(LATE):
                            send_bytes(0, 1, j)

                if (k, h) == (LATE, 1):
                    far_load.wait()

                    @pl.when(odd == 1)
                    def _():
                        e, m = _split(jnp.stack([x_far[...]] * 2))
                        via_bytes[2] = m[0]
                        detour(0, 0).start()
                        window, state = _encode_start(base, rank, _peak(e))
                        e = srl(e, I32(7))
                        codes, state = _encode_group(e, window, state)
                        pool, (level, _) = _encode_finish(window, state, tmp, (1, 1))
                        via_exps[2, 0] = codes[0]
                        via_exps[2, 1] = jnp.where(level < 2, pool[0][0], _level_bits(level))
                        levels[12] = level
                        detour(0, 1).start()

                        @pl.when(level == 2)
                        def _():
                            for j, v in enumerate(_plain(e[0, :8]) + _plain(e[0, 8:])):
                                via_exps[2, 2 + j] = v
                            detour(0, 2).start()

        for d in keep_loads[0]:
            d.start()
        encode_and_send(0, base, rank)
        for d in keep_loads[1]:
            d.start()
        for d in give_loads[-1]:
            d.wait()
        both = slice(None)
        each_64_rows(lambda r: stage(1, both, r, x_give[:, _rows(B + r, 64)]), then_send=1)

        @pl.when(p == 2)
        def _():
            for h in range(2):
                for k in range(2):
                    detour(h, k, incoming=True).wait_recv()
            header = [via_exps[h, 1, 0, 0] for h in range(2)]
            decode(via_exps, header, 1, (1,))
            for h in range(2):
                @pl.when(srl(header[h], I32(30)) == 2)
                def _():
                    detour(h, 2, incoming=True).wait_recv()
                    for j in range(2):
                        decoded[h, _pairs(16 * j, 16)] = _unplain(
                            [via_exps[h, 2 + 2 * j + k] for k in range(2)])

            v = _join(decoded[:, _pairs(0, ROUND)], via_bytes[:2]).astype(jnp.float32)
            stage(1, both, B - ROUND, x_give[:, pl.ds(Q - ROUND, ROUND)] + v)

        encode_and_send(1, *_pick_window(exps[:, :8]))

        for b in range(4):
            r0 = b % 2 * B
            wait_and_decode(b)
            wait_bytes(b, range(len(cuts[b])))
            if b < 2:
                for d in keep_loads[b]:
                    d.wait()
            if b == 1:
                @pl.when(p == 0)
                def _():
                    gone = _pairs(B - ROUND, ROUND)
                    bytes_in[1, :, gone] = jnp.zeros((2, ROUND // 2, N // 2), I32)
                    decoded[:, gone] = jnp.zeros((2, ROUND // 2, N), I32)

            def add(r):
                t = x_keep[:, _rows(r0 + r, 64)] + received(b, r, 64).astype(jnp.float32)
                if b < 2:
                    x_keep[:, _rows(r0 + r, 64)] = t
                else:
                    write(keep, r0 + r, t.astype(jnp.bfloat16))
                stage(b + 2, both, r, t)

            each_64_rows(add, then_send=b + 2)
            encode_and_send(b + 2, *_pick_window(exps[:, :8]))

        wait_and_decode(4)
        wait_bytes(4, range(len(cuts[4])))
        each_64_rows(lambda r: write(give, r, received(4, r, 64)))
        for b in range(5):
            wait_sent(b)

        @pl.when(odd == 1)
        def _():
            for k in range(2):
                detour(0, k).wait_send()
            pl.when(levels[12] == 2)(lambda: detour(0, 2).wait_send())

        wait_and_decode(5)
        for k, (r, n) in enumerate(cuts[5]):
            if k == len(cuts[5]) - 1:
                wait_sent(5)
            wait_bytes(5, [k])
            write(give, B + r, received(5, r, n))

    f32, vmem, dma = jnp.float32, pltpu.VMEM, pltpu.SemaphoreType.DMA
    return pl.pallas_call(
        body,
        out_shape=vmem((M, N), jnp.bfloat16),
        in_specs=[pl.BlockSpec(memory_space=pltpu.HBM)],
        out_specs=pl.BlockSpec(memory_space=vmem),
        scratch_shapes=[
            vmem((2, Q, N), f32),
            vmem((2, Q, N), f32),
            vmem((ROUND, N), f32),
            vmem((3, ROUND // 2, N // 2), I32),
            vmem((3, 6, 8, 128), I32),
            vmem((2, B // 2, N), I32),
            vmem((2, B // 2, 128), f32),
            vmem((2, B // 2, N), I32),
            vmem((2, 72, 128), I32),
            vmem((6, 2, B // 2, N // 2), I32),
            vmem((6, 2, B // 2, N // 2), I32),
            vmem((6, 2, sum(LEVELS[-1]), 8, 128), I32),
            vmem((6, 2, sum(LEVELS[-1]), 8, 128), I32),
            pltpu.SMEM((13,), I32),
            dma((2 * len(CUTS[0]) + 8,)),
            dma((2 * sem0[6] + 6,)),
            dma((2 * sem0[6] + 6,)),
            pltpu.SemaphoreType.REGULAR,
        ],
        compiler_params=pltpu.CompilerParams(collective_id=0, disable_semaphore_checks=True),
    )(x)
```

```python
import jax
import jax.numpy as jnp
from jax import lax
from jax.experimental import pallas as pl
from jax.experimental.pallas import tpu as pltpu

M, N = 2048, 512
Q = M // 4
B = Q // 2
GROUPS = B // 32

CUTS = (
    (16, 16, 32, 48, 64, 48, 32),
    (128, 128),
    (64, 128, 64),
    (128, 128),
    (128, 128),
    (64, 96, 64, 16, 16),
)
FRONT = (7, 1, 2, 1, 1, 1)
LATE = 3
ROUND = 32

POOL = (8, 9, 10, 11)
LEVELS = ((0, 11), (11, 1), (12, 22))
RUN = 6
HEADER = 14
STAND_IN = 20

I32 = jnp.int32
srl, sll = lax.shift_right_logical, lax.shift_left
VREGS = (2, 8, 128)


def _i(v):
    return I32(v - (1 << 32) if v >= (1 << 31) else v)


def _splat(v):
    return jnp.full(VREGS, _i(v), I32)


def _sublane():
    return lax.broadcasted_iota(I32, VREGS, 1)


def _header_bits():
    lane = lax.broadcasted_iota(I32, VREGS, 2)
    return jnp.where((_sublane() == 0) & (lane == 0), HEADER, 0)


def _with_header(pool, level, base, rank, stood_in):
    word = sll(level, I32(30)) | sll(base, I32(22)) | sll(rank, I32(19)) | sll(stood_in, I32(18))
    return jnp.where(level < 2, pool, 0) | jnp.where(_header_bits()[0] != 0, word, 0)


def _row(v, s):
    return jnp.broadcast_to(v[:, s : s + 1], VREGS)


def _both(v):
    return sll(v, I32(16)) | v


def _running_sum(v):
    for d in (1, 2, 4):
        v = v + jnp.where(_sublane() >= d, pltpu.roll(v, d, 1), 0)
    return v


def _rotate(v, n, up):
    for d in (1, 2, 4):
        v = jnp.where((n & d) != 0, pltpu.roll(v, 8 - d if up else d, 1), v)
    return v


def _shift_right(ws, n):
    rest = [srl(w, n) | sll(sll(u, I32(1)), n ^ 31) for u, w in zip(ws, ws[1:])]
    return [srl(ws[0], n)] + rest


def _shift_left(ws, n):
    rest = [sll(w, n) | srl(srl(u, I32(1)), n ^ 31) for w, u in zip(ws, ws[1:])]
    return rest + [sll(ws[-1], n)]


def _split(v):
    w = pltpu.bitcast(v.astype(jnp.bfloat16), I32)
    a, b = w[..., : N // 2], w[..., N // 2 :]
    rest = sll(b & _i(0x007F007F), I32(7)) | srl(b & _i(0x80008000), I32(1))
    return w & _i(0x7F807F80), (a & _i(0x807F807F)) | rest


def _join(e, m):
    b = (srl(m, I32(7)) & _i(0x007F007F)) | (sll(m, I32(1)) & _i(0x80008000))
    w = jnp.concatenate([m & _i(0x807F807F), b], axis=-1) | e
    return pltpu.bitcast(w, jnp.bfloat16)


def _pick_window(sample):
    t = sum(sample[..., j : j + 128] for j in range(0, N, 128))
    t = (srl(t, I32(16)) + (t & 0xFFFF)).astype(jnp.float32)
    t = jnp.sum(jnp.sum(t, axis=2, keepdims=True), axis=1, keepdims=True)
    mean = jnp.broadcast_to(t, VREGS) * (1.0 / (16 * N)) + 0.12
    whole = mean.astype(I32)
    rank = (7.9 - 6.3 * (mean - whole.astype(jnp.float32))).astype(I32)
    return jnp.clip(whole - 1, 0, 251), jnp.clip(rank, 1, 7)


def _peak(e):
    hi, lo = (lax.bitcast_convert_type(u, jnp.float32)
              for u in (srl(e, I32(1)), sll(e, I32(15))))
    t = jnp.maximum(hi, lo)
    t = jnp.maximum(t[..., :256], t[..., 256:])
    return jnp.maximum(t[..., :128], t[..., 128:])


def _encode_start(base, rank, peak):
    while peak.shape[1] > 8:
        n = peak.shape[1] // 2
        peak = jnp.maximum(peak[:, :n], peak[:, n:])
    top = srl(lax.bitcast_convert_type(peak, I32), I32(22))
    window = (base, rank, jnp.where(top > base + 4, top - base - 3, 1))
    return window, ([_splat(0)] * RUN, _splat(0), _splat(0))


def _replace(e, old, new):
    hi, lo = (jnp.where(v == old, new, v) for v in (srl(e, I32(16)), e & 0xFFFF))
    return sll(hi, I32(16)) | lo


def _plain(e):
    e = e[:, :256] | sll(e[:, 256:], I32(8))
    return e[:, :128], e[:, 128:]


def _unplain(vs):
    vs = [sll(v, I32(7)) for v in vs] + [srl(v, I32(1)) for v in vs]
    return jnp.concatenate(vs, axis=1) & _i(0x7F807F80)


def _encode_group(es, window, state):
    base, rank, above = window
    string, total, bad = state
    guard, top = _i(0x80008000), _splat(1 << 31)
    fence_lo, fence_hi = _both(base) | guard, guard - _both(base + 4)
    rank2, skip2, above2 = _both(rank), _both(rank - 1), _both(above)
    hi, lo = top, _splat(0)
    size = codes = _splat(0)
    for i in reversed(range(8)):
        e = es[:, i // 4 * 8 : i // 4 * 8 + 8, i % 4 * 128 : i % 4 * 128 + 128]
        t = fence_lo - e
        g = t & guard
        one = srl(g, I32(15))
        low = g - one
        g = (t - skip2) & guard
        skip = above2 & (g - srl(g, I32(15)))
        u = e + fence_hi
        g = u & guard
        high = g - srl(g, I32(15))
        n = (t & low) + one + skip + ((u + rank2) & high)
        codes = codes | sll(t & _i(0x00030003) & ~(low | high), I32(2 * i))
        n_hi = srl(n, I32(16))
        n = n_hi + (n & 0xFFFF)
        size, bad = size + n, bad | n
        lo = srl(lo, n) | sll(hi, n ^ 31)
        hi = srl(hi, n) | top | srl(top, n_hi)
    far = size >= 32
    string = [jnp.where(far, u, w) for u, w in zip([0] + string, string)]
    string = _shift_right(string, size & 31)
    string[0], string[1] = string[0] | hi, string[1] | sll(lo, I32(1))
    bad = bad | srl(size + 1, I32(1))
    return codes, (string, total + size, bad)


def _encode_finish(window, state, tmp, sizes):
    _, _, above = window
    string, total, bad = state
    total = total + above
    bad = (srl(bad | above, I32(5)) != 0) | (total > 32 * RUN)
    string = _shift_right(string, (above - 1) & 31)
    end = _running_sum(total + _header_bits())
    start = end - total
    string = _shift_right(string + [_splat(0)], start & 31) + [_splat(0)] * (7 - RUN)
    for j, w in enumerate(string):
        tmp[:, pl.ds(8 * j, 8)] = w
    first = srl(start, I32(5))
    pool = [_splat(0)] * sizes[1]
    for s in range(8):
        q = _row(first, s)
        w = _rotate(tmp[:, pl.ds(s, 8, stride=8)], q, up=False)
        at = srl(q + ((_sublane() - q) & 7), I32(3))
        pool = [v | jnp.where(at == j, w, 0) for j, v in enumerate(pool)]
    need = jnp.where(bad, 2000, end).astype(jnp.float32)
    need = [jnp.max(need[h]) for h in range(2)]
    level = [sum((v > 256 * n).astype(I32) for n in sizes) for v in need]
    return pool, level


def _decode_start(codes, pool, header, tmp):
    ones = _splat(1)
    for v in codes:
        ones = ones + lax.population_count(~(v | srl(v, I32(1))) & _i(0x55555555))
    before = _running_sum(ones) - ones
    pool = [srl(sll(pool[0], _header_bits()), _header_bits())] + pool[1:]
    first = passed = upto = _splat(0)
    for v in pool:
        seen = _running_sum(lax.population_count(v)) + upto
        for s in range(8):
            upto = _row(seen, s)
            ok = upto < before
            first, passed = jnp.where(ok, first + 1, first), jnp.where(ok, upto, passed)
    for s in range(8):
        q = _row(first, s)
        at = srl(q + ((_sublane() - q) & 7), I32(3))
        w = _splat(0)
        for j, v in enumerate(pool):
            w = jnp.where(at == j, v, w)
        tmp[:, pl.ds(8 * s, 8)] = _rotate(w, q, up=True)
    string = [tmp[:, pl.ds(j, 8, stride=8)] for j in range(RUN + 2)]
    left, w, skip = before - passed, string[0], _splat(0)
    for d in (16, 8, 4, 2, 1):
        c = lax.population_count(srl(w, I32(32 - d)))
        ok = c < left
        left, skip = jnp.where(ok, left - c, left), jnp.where(ok, skip + d, skip)
        w = jnp.where(ok, sll(w, I32(d)), w)
    opening = _sublane() == 0
    string = _shift_left(string, jnp.where(opening, _header_bits(), skip))[: RUN + 1]
    lead = lax.clz(jnp.where(opening, string[0], string[0] & _i(0x7FFFFFFF)) | 1)
    above = jnp.where(opening, lead + 1, lead)
    base, rank = srl(header, I32(22)) & 255, srl(header, I32(19)) & 7
    return (base, rank, above), _shift_left(string, lead)[:RUN]


def _decode_group(codes, window, string):
    base, rank, above = window
    roof = sll(_both(base + 4), I32(7))
    hi, lo = string[0], sll(string[0], I32(31)) | srl(string[1], I32(1))
    size, es = _splat(0), []
    for i in range(8):
        e, took = roof, []
        for at, to in ((16 + 2 * i, 23), (2 * i, 7)):
            code = srl(codes, I32(at)) & 3
            n = lax.clz(hi & _i(0x7FFFFFFF))
            u = rank - n
            drop = jnp.where(u > -above, jnp.where(u > 0, n + 3, u), n + (3 - above))
            e = e - sll(jnp.where(code == 0, drop, code), I32(to))
            took.append(jnp.where(code == 0, n, 0))
            hi = sll(hi, took[-1])
        n = took[0] + took[1]
        hi, lo = hi | srl(lo, n ^ 31), sll(lo, n)
        size = size + n
        es.append(e)
    far = size >= 32
    string = [jnp.where(far, u, w) for w, u in zip(string, string[1:] + [0])]
    es = [jnp.concatenate(es[i : i + 4], axis=2) for i in (0, 4)]
    return jnp.concatenate(es, axis=1), _shift_left(string, size & 31)


def _rows(r, n, unit=16):
    return pl.ds(r if isinstance(r, int) else pl.multiple_of(r, unit), n)


def _pairs(r, n):
    return _rows(r // 2, n // 2, 8)


def _plain_slot(j):
    return j + 1 + (j + 1 >= POOL[0]).astype(I32)


def pallas_dist_ar_i_i_m2048_n512_kernel(x: jax.Array):
    cuts = [[(sum(c[:k]), n) for k, n in enumerate(c)] for c in CUTS]
    sem0 = [sum(len(c) + len(LEVELS) for c in CUTS[:b]) for b in range(7)]

    def body(x_hbm, out, x_give, x_keep, x_far, via_bytes, via_exps, exps, peaks, decoded, tmp,
             bytes_out, bytes_in, exps_out, exps_in, levels, stood_in, ld, snd, rcv, ready):
        p = lax.axis_index("i")
        odd = p & 1
        half = [(p == 3).astype(I32) ^ h for h in range(2)]
        nbr = [p ^ (1 + 2 * v) for v in half]
        bit = [jnp.where(v == 0, (p ^ (p >> 1)) & 1, p >> 1) for v in half]
        keep = [(2 * half[h] + bit[h]) * Q for h in range(2)]
        give = [(2 * half[h] + 1 - bit[h]) * Q for h in range(2)]

        def signal(sem):
            for to in nbr[::-1]:
                pl.semaphore_signal(sem, 1, device_id=(to,), device_id_type=pl.DeviceIdType.MESH)

        def load(dst, base, k, r, n):
            return [
                pltpu.make_async_copy(
                    x_hbm.at[_rows(base[h] + r, n)], dst.at[h, pl.ds(r, n)], ld.at[2 * k + h])
                for h in range(2)
            ]

        def remote(src, dst, k, h, to, incoming):
            there = h if incoming else half[h] ^ (to == 3).astype(I32)
            return pltpu.make_async_remote_copy(
                src, dst(there), snd.at[2 * k + h], rcv.at[2 * k + there],
                device_id=(to,), device_id_type=pl.DeviceIdType.MESH)

        def block_copy(src, dst, b, h, part, k, incoming):
            return remote(src.at[b, h, part], lambda j: dst.at[b, j, part], sem0[b] + k,
                          h, nbr[h ^ (b // 2 == 1)], incoming)

        def with_copy(copy, act, h, incoming, has_rerouted_rows):
            if has_rerouted_rows:
                short = p == 0 if incoming else odd > h
                pl.when(short)(lambda: act(copy(1)))
                pl.when(~short)(lambda: act(copy(0)))
            else:
                act(copy(0))

        def with_exp_copy(b, h, level, act, incoming=False):
            def copy(omit):
                part = pl.ds(LEVELS[level][0] + omit, LEVELS[level][1] - omit)
                return block_copy(exps_out, exps_in, b, h, part, level, incoming)

            with_copy(copy, act, h, incoming, (b, level) == (1, 0))

        def with_byte_copy(b, h, k, act, incoming=False):
            def copy(omit):
                part = _pairs(cuts[b][k][0], cuts[b][k][1] - omit * ROUND)
                return block_copy(bytes_out, bytes_in, b, h, part, len(LEVELS) + k, incoming)

            with_copy(copy, act, h, incoming, (b, k) == (1, len(cuts[1]) - 1))

        def with_exp_copies(b, h, first, level, act, incoming=False):
            if first == 0:
                with_exp_copy(b, h, 0, act, incoming)
            for k in range(1, len(LEVELS)):
                pl.when(level >= k)(lambda: with_exp_copy(b, h, k, act, incoming))

        start = lambda d: d.start()
        sent = lambda d: d.wait_send()
        landed = lambda d: d.wait_recv()

        def detour(h, k, incoming=False):
            ref, part = ((via_bytes, slice(None)), (via_exps, pl.ds(0, 2)), (via_exps, pl.ds(2, 4)))[k]
            return remote(ref.at[2, part], lambda j: ref.at[j, part], sem0[6] + k, h, nbr[1], incoming)

        def send_bytes(b, h, k):
            with_byte_copy(b, h, k, start)

        def wait_bytes(b, ks):
            for k in ks:
                for h in range(2):
                    with_byte_copy(b, h, k, landed, incoming=True)

        def stage(b, hs, r, v):
            n = v.shape[1]
            e, m = _split(v)
            bytes_out[b, hs, _pairs(r, n)] = m
            exps[hs, _pairs(r, n)] = srl(e, I32(7))
            peaks[hs, _pairs(r, n)] = _peak(e)

        def each_64_rows(f, then_send=None):
            @pl.loop(0, B // 64, unroll=True)
            def _(t):
                f(t * 64)
                for k in range(FRONT[then_send] if then_send else 0):
                    @pl.when(t == sum(cuts[then_send][k]) // 64 - 1)
                    def _():
                        for h in range(2):
                            send_bytes(then_send, h, k)

        def stand_in(h, base):
            other = jnp.tile(base - STAND_IN, (B // 16, N // 128))
            e = exps[h]
            taken = jnp.where(other > 0, e ^ _replace(e, other, 0), 1)
            new = _replace(e, 0, other)
            found = [jnp.max(v.astype(jnp.float32)) > 0 for v in (taken, new ^ e)]

            @pl.when(~found[0] & found[1])
            def _():
                stood_in[h] = 1
                exps[h] = new

        def encode_and_send(b, base, rank):
            window, empty = _encode_start(base, rank, peaks[...])
            if b == 1:
                @pl.when(odd == 1)
                def _():
                    filler = _both(base[0] + 1)
                    exps[0, _pairs(B - ROUND, ROUND)] = jnp.tile(filler, (ROUND // 16, N // 128))

            def group(j, state):
                exps_out[b, :, j], state = _encode_group(
                    exps[:, _pairs(32 * (GROUPS - 1 - j), 32)], window, state)
                return state

            def encode():
                state = lax.fori_loop(0, GROUPS, group, empty, unroll=True)
                pool, level = _encode_finish(window, state, tmp, (3, 4))
                for at, v in zip(POOL[1:], pool[1:]):
                    exps_out[b, :, at] = v
                for h in range(2):
                    exps_out[b, h, POOL[0]] = _with_header(
                        pool[0][h], level[h], base[h], rank[h], stood_in[h])
                    levels[2 * b + h] = level[h]

            def attempt(done):
                encode()
                for h in range(2):
                    pl.when((done == 0) & (levels[2 * b + h] == 2))(lambda: stand_in(h, base[h]))
                again = (done == 0) & ((stood_in[0] | stood_in[1]) != 0)
                for h in range(2):
                    pl.when(again)(lambda: send_bytes(b, h, FRONT[b]))
                return jnp.where(again, 1, 2)

            for h in range(2):
                stood_in[h] = 0
            if b < 2:
                encode()
            else:
                lax.while_loop(lambda done: done < 2, attempt, I32(0))
            for h in range(2):
                level = levels[2 * b + h]

                @pl.when(level == 2)
                def _():
                    @pl.loop(0, B // 16)
                    def _(j):
                        for k, v in enumerate(_plain(exps[h, _pairs(16 * j, 16)])):
                            exps_out[b, h, _plain_slot(2 * j + k)] = v

                with_exp_copies(b, h, 0, level, start)
                for k in range(FRONT[b], len(cuts[b])):
                    if k == FRONT[b]:
                        pl.when((stood_in[0] | stood_in[1]) == 0)(lambda: send_bytes(b, h, k))
                    else:
                        send_bytes(b, h, k)

        def decode(msg, header, groups, pool):
            coded = [srl(v, I32(30)) < 2 for v in header]

            @pl.when(coded[0] | coded[1])
            def _():
                use = [jnp.where(coded[h], h, 1 - h) for h in range(2)]
                head = [jnp.where(coded[h], header[h], header[1 - h]) for h in range(2)]
                vreg = lambda at: jnp.stack([msg[use[h], at] for h in range(2)])
                window, string = _decode_start(
                    [vreg(j) for j in range(groups)], [vreg(at) for at in pool],
                    jnp.stack([jnp.full((8, 128), v, I32) for v in head]), tmp)

                def group(g, string):
                    decoded[:, _pairs(32 * g, 32)], string = _decode_group(
                        vreg(groups - 1 - g), window, string)
                    return string

                lax.fori_loop(0, groups, group, string, unroll=True)

        def wait_and_decode(b):
            for h in range(2):
                with_exp_copy(b, h, 0, landed, incoming=True)
            if b == 1:
                @pl.when(p == 0)
                def _():
                    exps_in[1, :, 0] = _splat(0xFFFFFFFF)

            header = [exps_in[b, h, POOL[0], 0, 0] for h in range(2)]
            level = [srl(v, I32(30)) for v in header]
            for h in range(2):
                @pl.when(level[h] == 0)
                def _():
                    exps_in[b, h, POOL[-1]] = jnp.zeros((8, 128), I32)

                with_exp_copies(b, h, 1, level[h], landed, incoming=True)

            decode(exps_in.at[b], header, GROUPS, POOL)
            for h in range(2):
                @pl.when(level[h] == 2)
                def _():
                    @pl.loop(0, B // 16)
                    def _(j):
                        decoded[h, _pairs(16 * j, 16)] = _unplain(
                            [exps_in[b, h, _plain_slot(2 * j + k)] for k in range(2)])

                if b >= 2:
                    @pl.when((srl(header[h], I32(18)) & 1) == 1)
                    def _():
                        other = (srl(header[h], I32(22)) & 255) - STAND_IN
                        decoded[h] = _replace(decoded[h], other * 128, 0)

        def received(b, r, n):
            return _join(decoded[:, _pairs(r, n)], bytes_in[b, :, _pairs(r, n)])

        def write(base, r, v):
            for h in range(2):
                out[_rows(base[h] + r, v.shape[1])] = v[h]

        def wait_sent(b):
            for h in range(2):
                for k in range(len(cuts[b])):
                    with_byte_copy(b, h, k, sent)
                with_exp_copies(b, h, 0, levels[2 * b + h], sent)

        give_loads = [load(x_give, give, k, r, n) for k, (r, n) in enumerate(cuts[0] + [(B, B)])]
        keep_loads = [load(x_keep, keep, len(give_loads) + k, k * B, B) for k in range(2)]
        far_load = pltpu.make_async_copy(
            x_hbm.at[_rows(give[0] + Q - ROUND, ROUND)], x_far, ld.at[2 * len(give_loads) + 4])

        barrier = pltpu.get_barrier_semaphore()
        pl.when(p != 2)(lambda: signal(barrier))
        give_loads[0][0].start()

        @pl.when(p == 2)
        def _():
            pl.semaphore_wait(barrier, 2)
            signal(ready)

        early = sum(give_loads[:-1], [])
        early.insert(2 * LATE + 2, far_load)
        for d in early[1:]:
            d.start()
        pl.when(p == 0)(lambda: pl.semaphore_wait(barrier, 2))
        pl.when(odd == 1)(lambda: pl.semaphore_wait(barrier, 1))

        for k, (r, n) in enumerate(cuts[0]):
            for h in range(2):
                give_loads[k][h].wait()
                stage(0, pl.ds(h, 1), r, x_give[pl.ds(h, 1), pl.ds(r, n)])
                if h == 0 or k >= LATE:
                    send_bytes(0, h, k)
                else:
                    pl.when(odd == 0)(lambda: send_bytes(0, 1, k))
                if k == 0:
                    give_loads[-1][h].start()
                if (k, h) == (LATE, 0):
                    base, rank = _pick_window(exps[:, :8])

                    @pl.when(odd == 1)
                    def _():
                        pl.semaphore_wait(ready, 1)
                        for j in range(LATE):
                            send_bytes(0, 1, j)

                if (k, h) == (LATE, 1):
                    far_load.wait()

                    @pl.when(odd == 1)
                    def _():
                        e, m = _split(jnp.stack([x_far[...]] * 2))
                        via_bytes[2] = m[0]
                        detour(0, 0).start()
                        window, state = _encode_start(base, rank, _peak(e))
                        e = srl(e, I32(7))
                        codes, state = _encode_group(e, window, state)
                        pool, (level, _) = _encode_finish(window, state, tmp, (1, 1))
                        via_exps[2, 0] = codes[0]
                        via_exps[2, 1] = _with_header(pool[0][0], level, base[0], rank[0], I32(0))
                        levels[12] = level
                        detour(0, 1).start()

                        @pl.when(level == 2)
                        def _():
                            for j, v in enumerate(_plain(e[0, :8]) + _plain(e[0, 8:])):
                                via_exps[2, 2 + j] = v
                            detour(0, 2).start()

        for d in keep_loads[0]:
            d.start()
        encode_and_send(0, base, rank)
        for d in keep_loads[1]:
            d.start()
        for d in give_loads[-1]:
            d.wait()
        both = slice(None)
        each_64_rows(lambda r: stage(1, both, r, x_give[:, _rows(B + r, 64)]), then_send=1)

        @pl.when(p == 2)
        def _():
            for h in range(2):
                for k in range(2):
                    detour(h, k, incoming=True).wait_recv()
            header = [via_exps[h, 1, 0, 0] for h in range(2)]
            decode(via_exps, header, 1, (1,))
            for h in range(2):
                @pl.when(srl(header[h], I32(30)) == 2)
                def _():
                    detour(h, 2, incoming=True).wait_recv()
                    for j in range(2):
                        decoded[h, _pairs(16 * j, 16)] = _unplain(
                            [via_exps[h, 2 + 2 * j + k] for k in range(2)])

            v = _join(decoded[:, _pairs(0, ROUND)], via_bytes[:2]).astype(jnp.float32)
            stage(1, both, B - ROUND, x_give[:, pl.ds(Q - ROUND, ROUND)] + v)

        encode_and_send(1, *_pick_window(exps[:, :8]))

        for b in range(4):
            r0 = b % 2 * B
            wait_and_decode(b)
            wait_bytes(b, range(len(cuts[b])))
            if b < 2:
                for d in keep_loads[b]:
                    d.wait()
            if b == 1:
                @pl.when(p == 0)
                def _():
                    gone = _pairs(B - ROUND, ROUND)
                    bytes_in[1, :, gone] = jnp.zeros((2, ROUND // 2, N // 2), I32)
                    decoded[:, gone] = jnp.zeros((2, ROUND // 2, N), I32)

            def add(r):
                t = x_keep[:, _rows(r0 + r, 64)] + received(b, r, 64).astype(jnp.float32)
                if b < 2:
                    x_keep[:, _rows(r0 + r, 64)] = t
                else:
                    write(keep, r0 + r, t.astype(jnp.bfloat16))
                stage(b + 2, both, r, t)

            each_64_rows(add, then_send=b + 2)
            encode_and_send(b + 2, *_pick_window(exps[:, :8]))

        wait_and_decode(4)
        wait_bytes(4, range(len(cuts[4])))
        each_64_rows(lambda r: write(give, r, received(4, r, 64)))
        for b in range(5):
            wait_sent(b)

        @pl.when(odd == 1)
        def _():
            for k in range(2):
                detour(0, k).wait_send()
            pl.when(levels[12] == 2)(lambda: detour(0, 2).wait_send())

        wait_and_decode(5)
        for k, (r, n) in enumerate(cuts[5]):
            if k == len(cuts[5]) - 1:
                wait_sent(5)
            wait_bytes(5, [k])
            write(give, B + r, received(5, r, n))

    f32, vmem, dma = jnp.float32, pltpu.VMEM, pltpu.SemaphoreType.DMA
    return pl.pallas_call(
        body,
        out_shape=vmem((M, N), jnp.bfloat16),
        in_specs=[pl.BlockSpec(memory_space=pltpu.HBM)],
        out_specs=pl.BlockSpec(memory_space=vmem),
        scratch_shapes=[
            vmem((2, Q, N), f32),
            vmem((2, Q, N), f32),
            vmem((ROUND, N), f32),
            vmem((3, ROUND // 2, N // 2), I32),
            vmem((3, 6, 8, 128), I32),
            vmem((2, B // 2, N), I32),
            vmem((2, B // 2, 128), f32),
            vmem((2, B // 2, N), I32),
            vmem((2, 72, 128), I32),
            vmem((6, 2, B // 2, N // 2), I32),
            vmem((6, 2, B // 2, N // 2), I32),
            vmem((6, 2, sum(LEVELS[-1]), 8, 128), I32),
            vmem((6, 2, sum(LEVELS[-1]), 8, 128), I32),
            pltpu.SMEM((13,), I32),
            pltpu.SMEM((2,), I32),
            dma((2 * len(CUTS[0]) + 8,)),
            dma((2 * sem0[6] + 6,)),
            dma((2 * sem0[6] + 6,)),
            pltpu.SemaphoreType.REGULAR,
        ],
        compiler_params=pltpu.CompilerParams(
            collective_id=0, disable_semaphore_checks=True, vmem_limit_bytes=32 * 2**20),
    )(x)
```
